```python
import numpy as np

kernel_name = "dist_sparse_attn_causalblk_htp_bs_b2_sq256_skv256_hq4_dh64"

def setup_inputs():
    x = np.random.randn(8, 256, 512).astype(np.float32)
    Wq = np.random.randn(512, 1024).astype(np.float32) * 0.02
    K_ext = np.random.randn(8, 256, 16, 64).astype(np.float32)
    V_ext = np.random.randn(8, 256, 16, 64).astype(np.float32)
    Wo = np.random.randn(1024, 512).astype(np.float32) * 0.02
    return {"x": x, "Wq": Wq, "K_ext": K_ext, "V_ext": V_ext, "Wo": Wo}

def reference(x, Wq, K_ext, V_ext, Wo):
    B, Sq, Skv, Hq, Dh = 8, 256, 256, 16, 64
    Q = (x @ Wq).reshape(B, Sq, Hq, Dh)
    qb = (np.arange(Sq) // 64)[:, None]
    kb = (np.arange(Skv) // 64)[None, :]
    mask = kb <= qb
    scores = np.einsum('bihd,bjhd->bhij', Q, K_ext).astype(np.float32) * 0.125
    scores = np.where(mask[None, None, :, :], scores, -1e9)
    scores_max = scores.max(axis=-1, keepdims=True)
    w = np.exp(scores - scores_max)
    row_keep = mask.any(axis=1)
    w_sum = np.where(row_keep[None, None, :, None], w.sum(axis=-1, keepdims=True), 1.0)
    w = w / w_sum
    w = np.where(row_keep[None, None, :, None], w, 0.0)
    ctx = np.einsum('bhij,bjhd->bihd', w, V_ext).reshape(B, Sq, Hq * Dh)
    return ctx @ Wo
```

```python
import contextlib

import jax
import jax.numpy as jnp
from jax import lax
from jax.experimental import pallas as pl
from jax.experimental.pallas import tpu as pltpu

bf16, f32 = jnp.bfloat16, jnp.float32
_MESH = pl.DeviceIdType.MESH
_NT = (((1,), (1,)), ((), ()))
_SCALE = 0.125 * 1.4426950408889634
SCOPES = False
OUT_DTYPE = bf16
ASYM = True


def _scope(name):
    return jax.named_scope(name) if SCOPES else contextlib.nullcontext()


def _dot(a, b):
    return jnp.dot(a, b, preferred_element_type=f32)


def _dot_nt(a, b):
    return lax.dot_general(a, b, _NT, preferred_element_type=f32)


def _low_lanes(rows):
    return lax.broadcasted_iota(jnp.int32, (rows, 128), 1) < 64


def _attention(qs, ks, vs):
    lo = _low_lanes(64)
    chains = [(u, t) for u in range(len(qs)) for t in (1, 0)]
    scores, res = {}, {}
    for u, t in chains:
        for j in (1, 0):
            blk = 2 * t + j
            q = qs[u][64 * blk:64 * blk + 64]
            h0, h1 = jnp.where(lo, q, 0.0), jnp.where(lo, 0.0, q)
            w = jnp.concatenate([h0, h1] if j == 0 else [h1, h0], axis=0)
            scores[u, t, j] = _dot_nt(ks[u][0:64 * (blk + 1), :], w.astype(bf16))
    for u, t in chains:
        nk = 128 * (t + 1)
        ps, inv = [], []
        for j in range(2):
            s = scores[u, t, j]
            p = jnp.exp2(s - jnp.max(s, axis=0, keepdims=True))
            inv.append(1.0 / jnp.sum(p, axis=0, keepdims=True))
            ps.append(pltpu.bitcast(p.astype(bf16), jnp.int32))
        p0 = jnp.concatenate([ps[0], jnp.zeros((32, 128), jnp.int32)], axis=0)
        lo_p, lo_1, lo_c = _low_lanes(nk // 2), _low_lanes(1), _low_lanes(32)
        top = _dot(vs[u][0:64, 0:nk], pltpu.bitcast(jnp.where(lo_p, p0, ps[1]), bf16))
        bot = _dot(vs[u][64:128, 0:nk], pltpu.bitcast(jnp.where(lo_p, ps[1], p0), bf16))
        top = top * jnp.where(lo_1, inv[0], inv[1])
        bot = bot * jnp.where(lo_1, inv[1], inv[0])
        c = pltpu.bitcast(jnp.concatenate([top, bot], axis=0).astype(bf16).T, jnp.int32)
        c = jnp.concatenate(
            [jnp.where(lo_c, c[0:32], c[32:64]), jnp.where(lo_c, c[32:64], c[0:32])], axis=0)
        res[u, t] = pltpu.bitcast(c, bf16)
    return [jnp.concatenate([res[u, 0], res[u, 1]], axis=0) for u in range(len(qs))]


_WQ_PIECES = ((0, 32), (32, 96), (128, 384))


def _body(x_hbm, wq_hbm, k_hbm, v_hbm, wo_hbm, o_ref,
          xf, wqf, wof, kf, vf, xb, wq, wo, kb, vb, ctx, acc,
          load_sem, send_sem, recv_sem, ready_sem):
    me = lax.axis_index("i")
    na, nb, nd = me ^ 1, 3 - me, me ^ 2
    odd = (me & 1) == 1
    barrier = pltpu.get_barrier_semaphore()

    def signal_neighbours(sem):
        for n in (na, nb):
            pl.semaphore_signal(sem, 1, device_id=(n,), device_id_type=_MESH)

    if ASYM:
        pl.when(me != 2)(lambda: signal_neighbours(barrier))
    else:
        signal_neighbours(barrier)

    n_load = [0]

    def load(src, dst):
        cp = pltpu.make_async_copy(src, dst, load_sem.at[n_load[0]])
        n_load[0] += 1
        cp.start()
        return cp

    wq_loads = [load(wq_hbm.at[pl.ds(r, n)], wqf.at[pl.ds(r, n)]) for r, n in _WQ_PIECES]
    x_load = load(x_hbm, xf)
    pair_of_slot = (2 * me, 2 * me + 1, 2 * na, 2 * nb + 1, 2 * na + 1, 2 * nb, 2 * nd, 2 * nd + 1)
    kv_loads = []
    for s, p in enumerate(pair_of_slot):
        rows = pl.ds(pl.multiple_of(128 * p, 128), 128)
        kv_loads.append((load(k_hbm.at[pl.ds(2 * me, 2), rows], kf.at[s]),
                         load(v_hbm.at[pl.ds(2 * me, 2), rows], vf.at[s])))
        if s == 1:
            wo_load = load(wo_hbm, wof)

    sends = []

    def send(src, dst, rsem, target):
        cp = pltpu.make_async_remote_copy(
            src, dst, send_sem.at[len(sends)], recv_sem.at[rsem],
            device_id=(target,), device_id_type=_MESH)
        cp.start()
        sends.append(cp)

    def wait_recv(dst, rsem):
        pltpu.make_async_remote_copy(
            dst, dst, send_sem.at[0], recv_sem.at[rsem],
            device_id=(me,), device_id_type=_MESH).wait_recv()

    with _scope("barrier"):
        if ASYM:
            pl.semaphore_wait(barrier, 2 - (me & 1))
            pl.when(me == 2)(lambda: signal_neighbours(ready_sem))
        else:
            pl.semaphore_wait(barrier, 2)

    s = (me == 3).astype(jnp.int32)
    first = jnp.where(me == 3, nb, na)
    second = jnp.where(me == 3, na, nb)
    with _scope("wq_prep"):
        for cp, (r, n) in zip(wq_loads, _WQ_PIECES):
            cp.wait()
            for h in range(2):
                wq[h, r:r + n, :] = wqf[r:r + n, 128 * h:128 * h + 128].astype(bf16)
            send(wq.at[s, pl.ds(r, n)], wq.at[2 + s, pl.ds(r, n)], s, first)
        send(wq.at[1 - s], wq.at[4 + s], 2 + s, first)
    with _scope("ready"):
        if ASYM:
            pl.when(odd)(lambda: pl.semaphore_wait(ready_sem, 1))
        send(wq.at[1 - s], wq.at[3 - s], 1 - s, second)
        send(wq.at[s], wq.at[5 - s], 3 - s, second)

    with _scope("x_prep"):
        x_load.wait()
        xb[...] = (xf[...].reshape(512, 512) * _SCALE).astype(bf16)

    def prep_kv(g):
        for sl in (2 * g, 2 * g + 1):
            kv_loads[sl][0].wait()
            kv_loads[sl][1].wait()
        for sl in (2 * g, 2 * g + 1):
            for b in range(2):
                kb[sl, b] = kf[sl, b].T.astype(bf16)
                vb[sl, b] = vf[sl, b].astype(bf16)

    def attend(g):
        q = _dot(xb[...], jnp.concatenate([wq[2 * g], wq[2 * g + 1]], axis=1))
        units = [(j, b) for j in range(2) for b in range(2)]
        outs = _attention([q[256 * b:256 * b + 256, 128 * j:128 * j + 128] for j, b in units],
                          [kb.at[2 * g + j, b] for j, b in units],
                          [vb.at[2 * g + j, b] for j, b in units])
        for (j, b), o in zip(units, outs):
            ctx[g, 256 * b:256 * b + 256, 128 * j:128 * j + 128] = o

    with _scope("kv0"):
        prep_kv(0)
    with _scope("wo_prep"):
        wo_load.wait()
        for n in range(4):
            wo[n, 0:256, :] = wof[:, 128 * n:128 * n + 128].astype(bf16)

    with _scope("wait_q1"):
        wait_recv(wq.at[2], 0)
        send(wq.at[2], wq.at[6], 4, nb)
        wait_recv(wq.at[3], 1)
        send(wq.at[3], wq.at[7], 5, na)

    def rows(slot):
        return pl.ds(128 * slot, 128)

    send(wo.at[:, rows(0)], wo.at[:, rows(2)], 6, na)
    send(wo.at[:, rows(1)], wo.at[:, rows(3)], 7, nb)
    send(wo.at[:, rows(1)], wo.at[:, rows(4)], 8, na)
    send(wo.at[:, rows(0)], wo.at[:, rows(5)], 9, nb)

    with _scope("attn0"):
        attend(0)
    with _scope("kv1"):
        prep_kv(1)
    with _scope("attn1"):
        attend(1)
    with _scope("kv2"):
        prep_kv(2)
        prep_kv(3)
    with _scope("wait_q2"):
        wait_recv(wq.at[4], 2)
        wait_recv(wq.at[5], 3)
    with _scope("attn2"):
        attend(2)
    with _scope("wait_q3"):
        wait_recv(wq.at[6], 4)
        wait_recv(wq.at[7], 5)
    with _scope("attn3"):
        attend(3)

    with _scope("wait_o1"):
        wait_recv(wo.at[:, rows(2)], 6)
        for n in range(4):
            send(wo.at[n, rows(2)], wo.at[n, rows(6)], 10 + n, nb)
        wait_recv(wo.at[:, rows(3)], 7)
        for n in range(4):
            send(wo.at[n, rows(3)], wo.at[n, rows(7)], 14 + n, na)

    def wo_cols(g):
        return jnp.concatenate([wo[n, 256 * g:256 * g + 256, :] for n in range(4)], axis=1)

    with _scope("out01"):
        acc[...] = _dot(ctx[0], wo_cols(0)) + _dot(ctx[1], wo_cols(1))
    with _scope("wait_o2"):
        wait_recv(wo.at[:, rows(4)], 8)
        wait_recv(wo.at[:, rows(5)], 9)
    with _scope("out2"):
        acc[...] += _dot(ctx[2], wo_cols(2))
    for n in range(4):
        if n == 3:
            for cp in sends[:-8]:
                cp.wait_send()
        with _scope(f"wait_o3_{n}"):
            wait_recv(wo.at[n, rows(6)], 10 + n)
            wait_recv(wo.at[n, rows(7)], 14 + n)
        with _scope(f"out3_{n}"):
            cols = slice(128 * n, 128 * n + 128)
            for b in range(2):
                r = slice(256 * b, 256 * b + 256)
                o_ref[b, :, cols] = (acc[r, cols] + _dot(ctx[3, r, :], wo[n, 768:1024, :])).astype(o_ref.dtype)
    for cp in sends[-8:]:
        cp.wait_send()


def pallas_dist_sparse_attn_causalblk_htp_bs_b2_sq256_skv256_hq4_dh64_kernel(x, Wq, K_ext, V_ext, Wo):
    kt = jnp.transpose(K_ext, (0, 2, 3, 1)).reshape(8, 1024, 256)
    vt = jnp.transpose(V_ext, (0, 2, 3, 1)).reshape(8, 1024, 256)
    return pl.pallas_call(
        _body,
        out_shape=jax.ShapeDtypeStruct(x.shape, OUT_DTYPE),
        in_specs=[pl.BlockSpec(memory_space=pltpu.HBM)] * 5,
        out_specs=pl.BlockSpec(memory_space=pltpu.VMEM),
        scratch_shapes=[
            pltpu.VMEM((2, 256, 512), f32),
            pltpu.VMEM((512, 256), f32),
            pltpu.VMEM((256, 512), f32),
            pltpu.VMEM((8, 2, 128, 256), f32),
            pltpu.VMEM((8, 2, 128, 256), f32),
            pltpu.VMEM((512, 512), bf16),
            pltpu.VMEM((8, 512, 128), bf16),
            pltpu.VMEM((4, 1024, 128), bf16),
            pltpu.VMEM((8, 2, 256, 128), bf16),
            pltpu.VMEM((8, 2, 128, 256), bf16),
            pltpu.VMEM((4, 512, 256), bf16),
            pltpu.VMEM((512, 512), f32),
            pltpu.SemaphoreType.DMA((21,)),
            pltpu.SemaphoreType.DMA((20,)),
            pltpu.SemaphoreType.DMA((18,)),
            pltpu.SemaphoreType.REGULAR,
        ],
        compiler_params=pltpu.CompilerParams(
            collective_id=0, vmem_limit_bytes=48 << 20,
            disable_bounds_checks=True, disable_semaphore_checks=True),
    )(x, Wq, kt, vt, Wo)
```

```python
import contextlib

import jax
import jax.numpy as jnp
import numpy as np
from jax import lax
from jax.experimental import pallas as pl
from jax.experimental.pallas import tpu as pltpu

bf16, f32, i32 = jnp.bfloat16, jnp.float32, jnp.int32
_MESH = pl.DeviceIdType.MESH
_NT = (((1,), (1,)), ((), ()))
_SCALE = 0.125 * 1.4426950408889634
SCOPES = False
OUT_DTYPE = bf16
INTERLEAVE = True
FWD1 = 1
FLAGS = {'XLA_TPU_FORCE_LP_LLO_SCHEDULER': True}


def _scope(name):
    return jax.named_scope(name) if SCOPES else contextlib.nullcontext()


def _k(v):
    return np.uint32(v & 0xFFFFFFFF).astype(np.int32) if isinstance(v, int) else v


def _and(a, b):
    return lax.bitwise_and(a, _k(b))


def _or(a, b):
    return b if a is None else lax.bitwise_or(a, _k(b))


def _add(a, b):
    return b if a is None else lax.add(a, _k(b))


def _sub(a, b):
    return lax.sub(_k(a), _k(b))


def _shl(a, n):
    return lax.shift_left(a, _k(n))


def _shr(a, n):
    return lax.shift_right_logical(a, _k(n))


def _move(a, n):
    return a if n == 0 else (_shl(a, n) if n > 0 else _shr(a, -n))


def _sel(m, a, b):
    a, b = (lax.full(m.shape, _k(v), i32) if isinstance(v, int) else v for v in (a, b))
    return lax.select(m, a, b)


def _words(x):
    return pltpu.bitcast(x.astype(bf16), i32)


def _halves(w):
    return pltpu.bitcast(w, bf16)


_SIGN_MANT = 0x807F807F
_EXPONENTS = 0x7F807F80
_PERIOD = 8
_STREAM_BITS = 56
_LOW, _SIDE, _FIELDS, _HIGH, _MSG = 0, 16, 18, 30, 46


def _swap_bytes(w, n):
    return _or(_shl(w, n), _shr(w, 32 - n))


def _pack_sign_mantissa(even, odd):
    return _or(_and(even, _SIGN_MANT), _swap_bytes(_and(odd, _SIGN_MANT), 8))


def _merge(low, exps):
    both = jnp.stack([low, _swap_bytes(low, 24)], axis=1)
    return _halves(_or(_and(both, _SIGN_MANT), exps).reshape(-1, 128))


def _encode_exponents(w_ref, msg_ref, raw_ref):
    exps = []
    top = None
    for j in range(16):
        w = w_ref[:, j]
        exps.append((_and(_shl(w, 16), 0x7F800000), _and(w, 0x7F800000)))
        m = lax.max(*(lax.bitcast_convert_type(e, f32) for e in exps[-1]))
        top = m if top is None else lax.max(top, m)
    top = lax.bitcast_convert_type(
        lax.max(lax.max(top[0], top[1]), lax.max(top[2], top[3])), i32)
    top4 = lax.broadcast_in_dim(top, (4, 8, 128), (1, 2))
    fields = [None] * 3
    runs = []
    for s in range(0, 16, _PERIOD):
        bits, zeros = lax.full((4, 8, 128), 0, i32), None
        for j in reversed(range(s, s + _PERIOD)):
            f = None
            for e in reversed(exps[j]):
                depth = _shr(_sub(top4, e), 23)
                deep = lax.gt(depth, _k(6))
                capped = _sel(deep, 7, depth)
                z = _sub(depth, capped)
                bits = _shr(_sel(deep, _or(_shr(bits, 1), 1 << 31), bits), _and(z, 31))
                zeros = _add(zeros, z)
                f = capped if f is None else _or(_shl(f, 16), capped)
            if j < 15:
                fields[j // 5] = _or(fields[j // 5], _move(f, 3 * (j % 5)))
            else:
                for k in range(3):
                    fields[k] = _or(fields[k], _shl(_and(f, 0x10001 << k), 15 - k))
        runs.append((bits, _add(zeros, lax.population_count(bits))))
    for k in range(3):
        msg_ref[_FIELDS + 4 * k:_FIELDS + 4 * k + 4] = fields[k]
    w0 = w1 = total = wide = None
    for blk in reversed(range(4)):
        for bits, n in reversed(runs):
            bits, n = bits[blk], n[blk]
            total, wide = _add(total, n), _or(wide, n)
            if w0 is None:
                w0, w1 = bits, lax.full((8, 128), 0, i32)
            else:
                n = _and(n, 31)
                w1 = _or(_shr(w1, n), _shl(_add(w0, w0), _sub(31, n)))
                w0 = _or(_shr(w0, n), bits)
    msg_ref[_SIDE] = w0
    msg_ref[_SIDE + 1] = _or(_and(w1, -2 << 8), _shr(top, 23))
    too_long = lax.bitwise_or(lax.gt(total, _k(_STREAM_BITS - 1)), lax.gt(wide, _k(31)))
    need_raw = jnp.max(jnp.where(too_long, 1.0, 0.0)) > 0.0

    @pl.when(need_raw)
    def _():
        msg_ref[_SIDE + 1] = lax.full((8, 128), 1 << 8, i32)
        msg_ref[_FIELDS:_HIGH] = lax.full((12, 8, 128), 0, i32)
        w = w_ref[...].reshape(32, 2, 8, 128)
        raw_ref[...] = _or(_and(w[:, 0], _EXPONENTS), _swap_bytes(_and(w[:, 1], _EXPONENTS), 8))

    return need_raw


def _sent_raw(msg_ref):
    return (msg_ref[_SIDE + 1][0, 0] & (1 << 8)) != 0


def _decode_exponents(msg_ref, out_ref):
    w0, w1 = msg_ref[:, _SIDE], msg_ref[:, _SIDE + 1]
    top = _and(w1, 0xFF)
    base = _or(_shl(top, 7), _shl(top, 23))
    for i in range(64):
        blk, j = divmod(i, 16)
        if i % _PERIOD == 0:
            if i:
                left = lax.clz(_and(bits, _sub(0, bits)))
                used = _sub(31, left)
                w0 = _or(_shl(w0, used), _shr(_shr(w1, 1), left))
                w1 = _shl(w1, used)
            bits = _or(w0, 1)
        if j < 15:
            f = _move(msg_ref[:, _FIELDS + 4 * (j // 5) + blk], 7 - 3 * (j % 5))
        else:
            f = None
            for k in range(3):
                f = _or(f, _shr(_and(msg_ref[:, _FIELDS + 4 * k + blk], 0x80008000), 8 - k))
        out = base
        for pos in (7, 23):
            capped = _and(f, 7 << pos)
            deep = lax.eq(capped, _k(7 << pos))
            z = lax.clz(bits)
            bits = _sel(deep, _shl(_add(bits, bits), z), bits)
            out = _sub(_sub(out, capped), _sel(deep, _shl(z, pos), 0))
        out_ref[:, i // 2, i % 2] = out
        yield


def _take_raw(raw_ref, out_ref):
    r = raw_ref[...]
    out_ref[:, 0] = _and(r, _EXPONENTS)
    out_ref[:, 1] = _and(_swap_bytes(r, 24), _EXPONENTS)


class _Filler:
    def __init__(self, *jobs):
        self.jobs = list(jobs)

    def emit(self, n):
        if not INTERLEAVE:
            return
        for job in self.jobs:
            for _ in range(n):
                next(job, None)

    def finish(self):
        for job in self.jobs:
            for _ in job:
                pass


def _dot(a, b):
    return jnp.dot(a, b, preferred_element_type=f32)


def _dot_nt(a, b):
    return lax.dot_general(a, b, _NT, preferred_element_type=f32)


def _low_lanes(rows):
    return lax.broadcasted_iota(i32, (rows, 128), 1) < 64


def _scores(q, k_ref, row, t):
    lo = _low_lanes(32)
    out = [None, None]
    for j in (1, 0):
        blk = 2 * t + j
        qq = q[32 * blk:32 * blk + 32]
        h0, h1 = _sel(lo, qq, 0), _sel(lo, 0, qq)
        w = lax.concatenate([h0, h1] if j == 0 else [h1, h0], 0)
        out[j] = _dot_nt(_halves(k_ref[row:row + 32 * (blk + 1), :]), _halves(w))
    return out


def _context(scores, v_ref, row, t):
    nk = 128 * (t + 1)
    ps, inv = [], []
    for s in scores:
        p = lax.exp2(s - jnp.max(s, axis=0, keepdims=True))
        total = jnp.sum(p, axis=0, keepdims=True)
        inv.append(1.0 / total)
        ps.append(p)
    both = _words(lax.concatenate([ps[0], ps[1][:nk - 64]], 1))
    last = _words(lax.concatenate([ps[1][nk - 64:nk - 32], ps[1][nk - 32:]], 1))
    p0 = lax.concatenate([both[:, :128], lax.full((32, 128), 0, i32)], 0)
    p1 = lax.concatenate([both[:, 128:], last[:, :128], last[:, 128:]], 0)
    lo, lo_p, lo_1 = _low_lanes(32), _low_lanes(nk // 2), _low_lanes(1)
    top = _dot(_halves(v_ref[row:row + 32, 0:nk]), _halves(_sel(lo_p, p0, p1)))
    bot = _dot(_halves(v_ref[row + 32:row + 64, 0:nk]), _halves(_sel(lo_p, p1, p0)))
    top = top * lax.select(lo_1, inv[0], inv[1])
    bot = bot * lax.select(lo_1, inv[1], inv[0])
    c = pltpu.bitcast(lax.concatenate([top, bot], 0).astype(bf16).T, i32)
    return lax.concatenate([_sel(lo, c[0:32], c[32:64]), _sel(lo, c[32:64], c[0:32])], 0)


_WQ_PIECES = ((0, 2), (2, 6), (8, 8))


def _body(x_hbm, wq_hbm, k_hbm, v_hbm, wo_hbm, o_ref,
          xf, wqf, wof, kf, vf, xb, wq, wo, kb, vb, qb, ctx, acc,
          mq, mo, rq, ro, eq_near, eq_far, eo_near, eo_far,
          load_sem, send_sem, recv_sem, ready_sem):
    me = lax.axis_index("i")
    na, nb, nd = me ^ 1, 3 - me, me ^ 2
    barrier = pltpu.get_barrier_semaphore()

    def signal_neighbours(sem):
        for n in (na, nb):
            pl.semaphore_signal(sem, 1, device_id=(n,), device_id_type=_MESH)

    n_load = [0]

    def load(src, dst):
        cp = pltpu.make_async_copy(src, dst, load_sem.at[n_load[0]])
        n_load[0] += 1
        cp.start()
        return cp

    s = (me == 3).astype(i32)
    first, second = jnp.where(me == 3, nb, na), jnp.where(me == 3, na, nb)

    def wq_cols(h):
        return pl.ds(pl.multiple_of(128 * h, 128), 128)

    wq_loads = [load(wq_hbm.at[pl.ds(32 * r, 32 * n), wq_cols(s)], wqf.at[0, pl.ds(32 * r, 32 * n)])
                for r, n in _WQ_PIECES]
    pl.when(me != 2)(lambda: signal_neighbours(barrier))
    wq_rest = load(wq_hbm.at[:, wq_cols(1 - s)], wqf.at[1])
    wo_load = load(wo_hbm, wof)
    x_loads = [load(x_hbm.at[b], xf.at[pl.ds(256 * b, 256)]) for b in range(2)]
    pair_of_slot = (2 * me, 2 * me + 1, 2 * na, 2 * nb + 1, 2 * na + 1, 2 * nb, 2 * nd, 2 * nd + 1)
    k_loads, v_loads = [], []

    def load_kv(g):
        for hbm, buf, loads in ((k_hbm, kf, k_loads), (v_hbm, vf, v_loads)):
            loads.append([
                load(hbm.at[2 * me + b, pl.ds(pl.multiple_of(128 * pair_of_slot[2 * g + j], 128), 128)],
                     buf.at[pl.ds(128 * (4 * g + 2 * b + j), 128)])
                for b in range(2) for j in range(2)])

    recv_ids = {}

    def remote(src, dst, ssem, rsem, target):
        return pltpu.make_async_remote_copy(
            src, dst, send_sem.at[ssem], recv_sem.at[rsem],
            device_id=(target,), device_id_type=_MESH)

    def recv_id(name, c):
        return 2 * recv_ids.setdefault(name, len(recv_ids)) + c

    def send(buf, src, dst, start, size, rsem, target, raw=False):
        rows = pl.ds(start, size)
        cp = remote(buf.at[src, rows], buf.at[dst, rows], 2 if raw else int(buf is mo), rsem, target)
        cp.start()
        if raw:
            cp.wait_send()

    def wait_recv(buf, slot, start, size, rsem):
        dst = buf.at[slot, pl.ds(start, size)]
        remote(dst, dst, 0, rsem, me).wait_recv()

    parts = {
        "q_first": (mq, (_LOW, _HIGH), 16), "q_exp": (mq, (_SIDE, _SIDE), 14),
        "q_second": (mq, (_HIGH, _LOW), 16), "o_exp": (mo, (_SIDE, _SIDE), 14),
        "q_raw": (rq, (0, 0), 32), "o_raw": (ro, (0, 0), 32),
        "far_q_exp": (mq, (_SIDE, _SIDE + 7), 7), "far_q": (mq, (_LOW, _HIGH), 16),
        "far_o_exp": (mo, (_SIDE, _SIDE + 7), 7),
        "far_q_raw": (rq, (0, 16), 16), "far_o_raw": (ro, (0, 16), 16),
    }
    for n in range(4):
        parts["o_first", n] = (mo, (_LOW + 4 * n, _HIGH + 4 * n), 4)
        parts["o_second", n] = (mo, (_HIGH + 4 * n, _LOW + 4 * n), 4)
        parts["far_o", n] = parts["o_first", n]

    def send_own(name, raw=False):
        buf, starts, size = parts[name]
        for c, target in ((0, na), (1, nb)):
            send(buf, 3, c, starts[c], size, recv_id(name, c), target, raw)

    def wait_near(name, which=(0, 1)):
        buf, starts, size = parts[name]
        for c in which:
            wait_recv(buf, c, starts[c], size, recv_id(name, c))

    def forward(name, which=(0, 1), raw=False):
        buf, starts, size = parts[name]
        for c in which:
            send(buf, c, 2, starts[c], size, recv_id(name, c), (nb, na)[c], raw)

    def wait_far(name):
        buf, starts, size = parts[name]
        for c in range(2):
            wait_recv(buf, 2, starts[c], size, recv_id(name, c))

    def near_raw(name, msg, raw, exps):
        flags = [_sent_raw(msg.at[c]) for c in range(2)]
        for c, flag in enumerate(flags):
            @pl.when(flag)
            def _():
                wait_near(name, (c,))
                forward("far_" + name, (c,), True)
                _take_raw(raw.at[c], exps.at[c])

    def far_raw(name, msg, raw, exps):
        @pl.when(_sent_raw(msg.at[2]))
        def _():
            wait_far(name)
            _take_raw(raw.at[2], exps.at[0])

    def split_wq(src, h, r, n):
        w = _words(wqf[src, 32 * r:32 * (r + n), :]).reshape(n, 2, 8, 128)
        mq[3, pl.ds(_HIGH * h + r, n)] = _pack_sign_mantissa(w[:, 0], w[:, 1])
        for c in range(r // 8, (r + n + 7) // 8):
            lo, hi = max(r, 8 * c), min(r + n, 8 * c + 8)
            wq[2 * h + c, 2 * (lo - 8 * c):2 * (hi - 8 * c)] = w[lo - r:hi - r].reshape(-1, 8, 128)

    def wait_all(copies):
        for cp in copies:
            cp.wait()

    def prep_k(g):
        for u in range(4 * g, 4 * g + 4):
            kb[128 * u:128 * u + 128] = pltpu.bitcast(kf[128 * u:128 * u + 128].astype(bf16).T, i32)
            yield

    def prep_v(g):
        for u in range(4 * g, 4 * g + 4):
            vb[64 * u:64 * u + 64] = _words(vf[128 * u:128 * u + 128])
            yield

    source = {1: ((0, 0), (1, 1)), 2: ((0, 1), (1, 0)), 3: ((2, 0), (2, 1))}

    def wq_of(g):
        if g == 0:
            return lax.concatenate([_halves(wq[2 * h:2 * h + 2].reshape(256, 128)) for h in range(2)], 1)
        return lax.concatenate(
            [_merge(mq[c, pl.ds(_HIGH * h, 16)], (eq_far if c == 2 else eq_near)[c % 2, pl.ds(16 * h, 16)])
             for c, h in source[g]], 1)

    def wo_of(g, n):
        if g == 0:
            return _halves(lax.concatenate(
                [wo[2 * h + n // 2, 8 * (n % 2):8 * (n % 2) + 8].reshape(64, 128) for h in range(2)], 0))
        return lax.concatenate(
            [_merge(mo[c, pl.ds(_HIGH * h + 4 * n, 4)],
                    (eo_far if c == 2 else eo_near)[c % 2, pl.ds(16 * h + 4 * n, 4)])
             for c, h in source[g]], 0)

    def project_q(g, filler, batches=(0, 1)):
        w = wq_of(g)
        for b in batches:
            qb[128 * b:128 * b + 128, 256 * g:256 * g + 256] = _words(
                _dot(_halves(xb[128 * b:128 * b + 128]), w))
            filler.emit(32)
        filler.finish()

    def scores(g, batches=(0, 1)):
        out = []
        for b in batches:
            for j in range(2):
                q = qb[128 * b:128 * b + 128, 256 * g + 128 * j:256 * g + 128 * j + 128]
                for t in (1, 0):
                    out.append((g, b, j, t, _scores(q, kb, 128 * (4 * g + 2 * b + j), t)))
        return out

    def contexts(sc):
        for g, b, j, t, s_ in sc:
            ctx[128 * b + 64 * t:128 * b + 64 * t + 64, 256 * g + 128 * j:256 * g + 128 * j + 128] = (
                _context(s_, vb, 64 * (4 * g + 2 * b + j), t))

    def project_out(groups, tiles, filler, batches=(0, 1)):
        w = lax.concatenate([lax.concatenate([wo_of(g, n) for g in groups], 0) for n in tiles], 1)
        cols = slice(128 * tiles[0], 128 * tiles[-1] + 128)
        for b in batches:
            rows = slice(256 * b, 256 * b + 256)
            r = _dot(_halves(ctx[128 * b:128 * b + 128, 256 * groups[0]:256 * groups[-1] + 256]), w)
            if groups[0]:
                r = acc[rows, cols] + r
            if groups[-1] == 3:
                o_ref[rows, cols] = r.astype(o_ref.dtype)
            else:
                acc[rows, cols] = r
            filler.emit(32)
        filler.finish()

    root = me == 0
    with _scope("barrier"):
        pl.when(me != 0)(lambda: pl.semaphore_wait(barrier, 2 - (me & 1)))
        pl.when(me == 2)(lambda: signal_neighbours(ready_sem))
    with _scope("wq_low"):
        for cp, (r, n) in zip(wq_loads, _WQ_PIECES):
            cp.wait()
            split_wq(0, s, r, n)
            pl.when(me != 0)(
                lambda: send(mq, 3, s, _HIGH * s + r, n, recv_id("q_first", s), first))
        wq_rest.wait()
        split_wq(1, 1 - s, 0, 16)
    with _scope("ready"):
        pl.when((me & 1) == 1)(lambda: pl.semaphore_wait(ready_sem, 1))
        pl.when(me != 0)(
            lambda: send(mq, 3, 1 - s, _HIGH * (1 - s), 16, recv_id("q_first", 1 - s), second))
    with _scope("wq_enc"):
        load_kv(0)
        raw_q = _encode_exponents(wq, mq.at[3], rq.at[3])
    with _scope("barrier0"):
        @pl.when(root)
        def _():
            pl.semaphore_wait(barrier, 2)
            send_own("q_first")
        send_own("q_exp")
        pl.when(raw_q)(lambda: send_own("q_raw", True))
        send_own("q_second")
    with _scope("wo_wait"):
        wo_load.wait()
    with _scope("wo_enc"):
        for h in range(2):
            words = _words(wof[128 * h:128 * h + 128, :])
            for n in range(4):
                w = words[:, 128 * n:128 * n + 128].reshape(4, 2, 8, 128)
                mo[3, pl.ds(_HIGH * h + 4 * n, 4)] = _pack_sign_mantissa(w[:, 0], w[:, 1])
                wo[2 * h + n // 2, 8 * (n % 2):8 * (n % 2) + 8] = w.reshape(8, 8, 128)
        raw_o = _encode_exponents(wo, mo.at[3], ro.at[3])
        send_own("o_exp")
        pl.when(raw_o)(lambda: send_own("o_raw", True))
    for b in range(2):
        with _scope("x_wait"):
            x_loads[b].wait()
        with _scope("q0"):
            xb[128 * b:128 * b + 128] = _words(xf[256 * b:256 * b + 256] * _SCALE)
            project_q(0, _Filler(), (b,))
    with _scope("k0_wait"):
        load_kv(1)
        wait_all(k_loads[0])
    with _scope("attn0"):
        _Filler(prep_k(0)).finish()
        sc = scores(0)
        wait_all(v_loads[0])
        _Filler(prep_v(0)).finish()
        contexts(sc)
    with _scope("w1"):
        load_kv(2)
        wait_near("q_first")
        wait_near("q_exp")
        forward("far_q_exp")
        forward("far_q")
        for n in range(4):
            send_own(("o_first", n))
    with _scope("out0"):
        project_out((0,), (0, 1, 2, 3), _Filler(_decode_exponents(mq.at[0:2], eq_near)))
        near_raw("q_raw", mq, rq, eq_near)
    with _scope("w2"):
        load_kv(3)
        wait_all(k_loads[1] + v_loads[1])
    with _scope("q1"):
        project_q(1, _Filler(prep_k(1), prep_v(1)))
    with _scope("w3"):
        wait_near("q_second")
        wait_all(k_loads[2])
    with _scope("attn1q2"):
        sc = scores(1)
        project_q(2, _Filler(prep_k(2)), (0,))
        contexts(sc)
        project_q(2, _Filler(), (1,))
    with _scope("w4"):
        wait_near("o_exp")
        forward("far_o_exp")
        for n in range(4):
            send_own(("o_second", n))
        wait_far("far_q_exp")
        wait_all(v_loads[2])
    with _scope("attn2"):
        sc = scores(2)
        _Filler(prep_v(2)).finish()
        contexts(sc)
        _Filler(_decode_exponents(mq.at[2:3], eq_far)).finish()
        far_raw("far_q_raw", mq, rq, eq_far)
    with _scope("w5"):
        wait_far("far_q")
        wait_all(k_loads[3] + v_loads[3])
        for n in range(FWD1):
            wait_near(("o_first", n))
            forward(("far_o", n))
    with _scope("q3"):
        project_q(3, _Filler(prep_k(3), prep_v(3), _decode_exponents(mo.at[0:2], eo_near)))
        near_raw("o_raw", mo, ro, eo_near)
    with _scope("w6"):
        for n in range(FWD1, 4):
            wait_near(("o_first", n))
            forward(("far_o", n))
    with _scope("attn3out1"):
        sc = scores(3)
        project_out((1,), (0, 1, 2, 3), _Filler(), (0,))
        contexts(sc)
        project_out((1,), (0, 1, 2, 3), _Filler(), (1,))
    with _scope("w8"):
        wait_far("far_o_exp")
        for n in range(3):
            wait_near(("o_second", n))
    with _scope("out2_012"):
        project_out((2,), (0, 1, 2), _Filler(_decode_exponents(mo.at[2:3], eo_far)))
        far_raw("far_o_raw", mo, ro, eo_far)
    with _scope("w"):
        wait_near(("o_second", 3))
        wait_far(("far_o", 0))
    with _scope("out2_3"):
        project_out((2,), (3,), _Filler())
        project_out((3,), (0,), _Filler())
    for n in range(1, 4):
        with _scope("w"):
            wait_far(("far_o", n))
        with _scope(f"out3_{n}"):
            project_out((3,), (n,), _Filler())
    for k, buf in enumerate((mq, mo)):
        remote(buf.at[0:3], buf.at[0:3], k, 0, me).wait_send()


def pallas_dist_sparse_attn_causalblk_htp_bs_b2_sq256_skv256_hq4_dh64_kernel(x, Wq, K_ext, V_ext, Wo):
    kt = jnp.transpose(K_ext, (0, 2, 3, 1)).reshape(8, 1024, 256)
    vt = jnp.transpose(V_ext, (0, 2, 3, 1)).reshape(8, 1024, 256)
    return pl.pallas_call(
        _body,
        out_shape=jax.ShapeDtypeStruct((512, 512), OUT_DTYPE),
        in_specs=[pl.BlockSpec(memory_space=pltpu.HBM)] * 5,
        out_specs=pl.BlockSpec(memory_space=pltpu.VMEM),
        scratch_shapes=[
            pltpu.VMEM((512, 512), f32),
            pltpu.VMEM((2, 512, 128), f32),
            pltpu.VMEM((256, 512), f32),
            pltpu.VMEM((2048, 256), f32),
            pltpu.VMEM((2048, 256), f32),
            pltpu.VMEM((256, 512), i32),
            pltpu.VMEM((4, 16, 8, 128), i32),
            pltpu.VMEM((4, 16, 8, 128), i32),
            pltpu.VMEM((2048, 128), i32),
            pltpu.VMEM((1024, 256), i32),
            pltpu.VMEM((256, 1024), i32),
            pltpu.VMEM((256, 1024), i32),
            pltpu.VMEM((512, 512), f32),
            pltpu.VMEM((4, _MSG, 8, 128), i32),
            pltpu.VMEM((4, _MSG, 8, 128), i32),
            pltpu.VMEM((4, 32, 8, 128), i32),
            pltpu.VMEM((4, 32, 8, 128), i32),
            pltpu.VMEM((2, 32, 2, 8, 128), i32),
            pltpu.VMEM((1, 32, 2, 8, 128), i32),
            pltpu.VMEM((2, 32, 2, 8, 128), i32),
            pltpu.VMEM((1, 32, 2, 8, 128), i32),
            pltpu.SemaphoreType.DMA((39,)),
            pltpu.SemaphoreType.DMA((3,)),
            pltpu.SemaphoreType.DMA((46,)),
            pltpu.SemaphoreType.REGULAR,
        ],
        compiler_params=pltpu.CompilerParams(
            collective_id=0, flags=FLAGS, vmem_limit_bytes=48 << 20,
            disable_bounds_checks=True, disable_semaphore_checks=True),
    )(x, Wq, kt, vt, Wo).reshape(x.shape)
```

```python
import jax
import jax.numpy as jnp
import numpy as np
from jax import lax
from jax.experimental import pallas as pl
from jax.experimental.pallas import tpu as pltpu

bf16, f32, i32 = jnp.bfloat16, jnp.float32, jnp.int32
_MESH = pl.DeviceIdType.MESH
_SCORE_SCALE = 0.125 * 1.4426950408889634


def _const(v):
    return np.uint32(v & 0xFFFFFFFF).astype(np.int32) if isinstance(v, int) else v


def _and(a, b):
    return lax.bitwise_and(a, _const(b))


def _or(a, b):
    return b if a is None else lax.bitwise_or(a, _const(b))


def _add(a, b):
    return b if a is None else lax.add(a, _const(b))


def _sub(a, b):
    return lax.sub(_const(a), _const(b))


def _shl(a, n):
    return lax.shift_left(_const(a), _const(n))


def _shr(a, n):
    return lax.shift_right_logical(_const(a), _const(n))


def _move(a, n):
    return a if n == 0 else (_shl(a, n) if n > 0 else _shr(a, -n))


def _rotl(a, n):
    return _or(_shl(a, n), _shr(a, 32 - n))


def _pick(mask, a, b):
    a, b = (lax.full(mask.shape, _const(v), i32) if isinstance(v, int) else v for v in (a, b))
    return lax.select(mask, a, b)


def _words(x):
    return pltpu.bitcast(x.astype(bf16), i32)


def _halves(w):
    return pltpu.bitcast(w, bf16)


_SIGN_MANTISSA = 0x807F807F
_EXPONENT = 0x7F807F80
_OWN_WORDS, _MAX_WORDS, _POOL_WORDS = 5, 9, 10
_HEAD = 8 * _OWN_WORDS
_POOL = _HEAD + 3
_STREAM_ROWS = _POOL + _POOL_WORDS


def _fuse(pairs, mask):
    return _or(_and(pairs[:, 0], mask), _rotl(_and(pairs[:, 1], mask), 8))


def _rebuild(low, coarse):
    out = []
    for k, bits in enumerate((low, _rotl(low, 24))):
        bits = _and(bits, _SIGN_MANTISSA)
        out.append(_or(_and(_sub(coarse[:, k], bits), _EXPONENT), bits))
    return lax.concatenate(out, 1).reshape(-1, 128)


def _choose_top(w_ref, half):
    peak = total = None
    for r in range(4 * half, 4 * half + 4):
        for j in (0, 4):
            w = w_ref[r, j:j + 4]
            m = lax.max(*(lax.bitcast_convert_type(_and(v, 0x3FFF8000), f32)
                          for v in (_shl(w, 15), _shr(w, 1))))
            peak = m if peak is None else lax.max(peak, m)
            total = _add(total, _and(_shr(w, 7), 0xFF00FF))
    peak = jnp.max(peak.reshape(32, 128), axis=0, keepdims=True)
    peak = _shr(lax.bitcast_convert_type(jnp.broadcast_to(peak, (8, 128)), i32), 15)
    total = _add(_and(total, 0xFFFF), _shr(total, 16)).reshape(32, 128).astype(f32)
    top = jnp.sum(total, axis=0, keepdims=True) * 0.25 + 469.0
    top = jnp.broadcast_to(top, (8, 128)).astype(i32)
    return _pick(lax.gt(peak, top), peak, top)


def _encode(w_ref, half, top, field_ref, stream):
    top = _or(_shl(top, 16), top)

    def run(r, stream):
        words, end, widest = stream
        fields = pos = b0 = b1 = None
        for j in range(8):
            gap = _sub(top, _and(w_ref[r, j], 0x7FFF7FFF))
            pair = None
            for depth, at in ((_and(_shr(gap, 7), 0x1FF), 2 * j), (_shr(gap, 23), 2 * j + 16)):
                deep = lax.gt(depth, _const(3))
                fields = _or(fields, _move(_pick(deep, 0, depth), at))
                n = _pick(deep, _sub(depth, _pick(lax.lt(depth, _const(7)), 3, 2)),
                          _pick(lax.eq(depth, _const(0)), 4, 0))
                pos, pair = _add(pos, n), _add(pair, n)
                stop, early = _shr(1 << 31, _and(pos, 31)), lax.lt(pos, _const(32))
                b0, b1 = _or(b0, _pick(early, stop, 0)), _or(b1, _pick(early, 0, stop))
            widest = _or(widest, pair)
        field_ref[r] = fields
        word, at = _shr(end, 5), _and(end, 31)
        back = _sub(31, at)
        parts = (_shr(b0, at), _or(_shr(b1, at), _shl(_add(b0, b0), back)), _shl(_add(b1, b1), back))
        here = [lax.eq(word, _const(i)) for i in range(_MAX_WORDS)]
        grown = []
        for i, w in enumerate(words):
            new = 0
            for k, part in enumerate(parts[:i + 1]):
                new = _pick(here[i - k], part, new)
            grown.append(_or(w, new))
        return tuple(grown), _add(end, pos), _or(widest, _shr(pos, 1))

    return lax.fori_loop(4 * half, 4 * half + 4, run, stream)


def _write_stream(tops, stream, ref):
    words, end, widest = stream
    for i in range(_OWN_WORDS):
        ref[8 * i:8 * i + 8] = words[i]
    extra = _sub(_shr(end, 5), _OWN_WORDS - 1)
    extra = _pick(lax.gt(extra, _const(0)), extra, 0)
    rows = [_add(lax.broadcasted_iota(i32, (8, 128), 0), 8 * i + _HEAD - _POOL) for i in range(2)]
    used = offsets = lax.full((8, 128), 0, i32)
    pool = [used, used]
    for s in range(8):
        offsets = _or(offsets, _move(_and(used, 15), 4 * s))
        ahead = [_sub(r, used) for r in rows]
        for k, word in enumerate(words[_OWN_WORDS:]):
            word = jnp.broadcast_to(word[s:s + 1], (8, 128))
            pool = [_pick(lax.eq(a, _const(k)), word, p) for a, p in zip(ahead, pool)]
        used = _add(used, jnp.broadcast_to(extra[s:s + 1], (8, 128)))
    heads = (_or(tops[0], _shl(tops[1], 16)), _or(tops[2], _shl(tops[3], 16)), offsets)
    for i, head in enumerate(heads):
        pool[0] = _pick(lax.eq(rows[0], _const(i + _HEAD - _POOL)), head, pool[0])
    ref[_HEAD:_HEAD + 8] = pool[0]
    ref[_HEAD + 8:_HEAD + 16] = pool[1]
    over = (widest > 31) | (end >= 32 * _MAX_WORDS) | (used > _POOL_WORDS)
    return jnp.max(jnp.where(over, 1.0, 0.0)) > 0.0


def _stream_row(stream_ref, i):
    return jnp.broadcast_to(stream_ref[:, i:i + 1, :], (stream_ref.shape[0], 8, 128))


def _open_stream(stream_ref):
    words = [stream_ref[:, 8 * i:8 * i + 8, :] for i in range(_OWN_WORDS)]
    sublane = lax.broadcasted_iota(i32, words[0].shape, 1)
    offset = _and(_shr(_stream_row(stream_ref, _HEAD + 2), _shl(sublane, 2)), 15)
    more = [-1] * (_MAX_WORDS - _OWN_WORDS)
    for i in range(_POOL_WORDS):
        mine = lax.eq(offset, _const(i))
        more = [_pick(mine, _stream_row(stream_ref, _POOL + i + k), m) if i + k < _POOL_WORDS else m
                for k, m in enumerate(more)]
    return tuple(words + more), lax.full(words[0].shape, 0, i32)


def _decode(top, field_ref, out_ref, first, last, state):
    base = _add(_or(_shl(top, 16), top), 0x80008000)

    def run(r, state):
        words, pos = state
        one, two = lax.gt(pos, _const(31)), lax.gt(pos, _const(63))
        words = words + (-1, -1)
        words = tuple(_pick(two, c, _pick(one, b, a)) for a, b, c in zip(words, words[1:], words[2:]))
        pos = _and(pos, 31)
        back = _sub(31, pos)
        w0, w1 = (_or(_shl(a, pos), _shr(_shr(b, 1), back)) for a, b in zip(words[:2], words[1:3]))
        fields = field_ref[:, r]
        for j in range(8):
            aligned, out, used = _move(fields, 7 - 2 * j), base, None
            for at in (7, 23):
                shallow = _and(aligned, 3 << at)
                escape = lax.eq(shallow, _const(0))
                w0 = _and(w0, 0x7FFFFFFF)
                n = _pick(escape, lax.clz(w0), 0)
                w0, used = _shl(w0, n), _add(used, n)
                deep = _shl(_add(n, _pick(lax.lt(n, _const(4)), 3, 2)), at)
                out = _sub(out, _pick(lax.bitwise_and(escape, lax.ne(n, _const(4))), deep, shallow))
            if j < 7:
                w0, w1 = _or(w0, _shr(_shr(w1, 1), _sub(31, used))), _shl(w1, used)
            pos = _add(pos, used)
            out_ref[:, 4 * r + j // 2, j % 2] = out
        return words, pos

    return lax.fori_loop(first, last, run, state, unroll=True)


def _dot(a, b):
    return jnp.dot(a, b, preferred_element_type=f32)


def _low_lanes(rows):
    return lax.broadcasted_iota(i32, (rows, 128), 1) < 64


def _scores(q, k_ref, row, tile):
    low, out = _low_lanes(32), [None, None]
    for j in (1, 0):
        block = 2 * tile + j
        qq = q[32 * block:32 * block + 32]
        heads = [_pick(low, qq, 0), _pick(low, 0, qq)]
        out[j] = lax.dot_general(
            _halves(k_ref[row:row + 32 * (block + 1), :]),
            _halves(lax.concatenate(heads[::1 - 2 * j], 0)),
            (((1,), (1,)), ((), ())), preferred_element_type=f32)
    return out


def _context(scores, v_ref, row, tile):
    keys = 128 * (tile + 1)
    p, inv = [], []
    for s in scores:
        p.append(lax.exp2(s - jnp.max(s, axis=0, keepdims=True)))
        inv.append(1.0 / jnp.sum(p[-1], axis=0, keepdims=True))
    p[0] = lax.concatenate([p[0], lax.full((64, 128), 0.0, f32)], 0)
    low, low_row = _low_lanes(keys), _low_lanes(1)
    heads = [(lax.select(low, p[h], p[1 - h]).astype(bf16), lax.select(low_row, inv[h], inv[1 - h]))
             for h in range(2)]
    return lax.concatenate(
        [_dot(_halves(v_ref[row + 32 * h:row + 32 * h + 32, 0:keys]), weights) * scale
         for h, (weights, scale) in enumerate(heads)], 0)


def _by_query(context):
    c, low = pltpu.bitcast(context.astype(bf16).T, i32), _low_lanes(32)
    return lax.concatenate([_pick(low, c[0:32], c[32:64]), _pick(low, c[32:64], c[0:32])], 0)


_FAR, _OWN = 2, 3
_LOW_Q, _LOW_O, _FIELDS_Q, _FIELDS_O, _STREAM, _PLAIN = range(6)
_PARTS = {
    "q0": (_LOW_Q, (0, 16), (0, 16)),
    "q1 head": (_LOW_Q, (16, 2), (16, 2)),
    "q1 rest": (_LOW_Q, (18, 14), (18, 14)),
    "far q0": (_LOW_Q, (0, 8), (8, 8)),
    "far q1": (_LOW_Q, (16, 8), (24, 8)),
    "q fields": (_FIELDS_Q, (0, 8), (0, 8)),
    "far q fields": (_FIELDS_Q, (0, 4), (4, 4)),
    "o fields 0": (_FIELDS_O, (0, 4), (0, 4)),
    "o fields 1": (_FIELDS_O, (4, 4), (4, 4)),
    "far o fields": (_FIELDS_O, (0, 4), (4, 4)),
    "stream": (_STREAM, (0, _STREAM_ROWS), (0, _STREAM_ROWS)),
    "far stream": (_STREAM, (0, 26), (26, _STREAM_ROWS - 26)),
    "o head": (_LOW_O, (0, 2), (16, 2)),
    "o01": (_LOW_O, (2, 6), (18, 6)),
    "o2": (_LOW_O, (8, 4), (24, 4)),
    "o3": (_LOW_O, (12, 4), (28, 4)),
    "other o01": (_LOW_O, (16, 8), (0, 8)),
    "other o23": (_LOW_O, (24, 8), (8, 8)),
    "far o01": (_LOW_O, (0, 8), (16, 8)),
    "far o2": (_LOW_O, (8, 4), (24, 4)),
    "far o3": (_LOW_O, (12, 4), (28, 4)),
    "plain": (_PLAIN, (0, 2), (0, 2)),
    "far plain": (_PLAIN, (0, 1), (1, 1)),
}
_FIRST_PIECES = ((0, 2), (2, 6), (8, 8))
_Q_GROUPS = (None, ((0, 0), (1, 0)), ((0, 1), (1, 1)), ((_FAR, 0), (_FAR, 1)))
_O_GROUPS = (None, ((0, 0), (1, 1)), ((0, 1), (1, 0)), ((_FAR, 0), (_FAR, 1)))
_CONTEXT_COLUMN = (0, 1, 2, 5, 4, 3, 6, 7)


def _body(x_hbm, wq_hbm, k_hbm, v_hbm, wo_hbm, out_ref,
          x_f32, wq_f32, wo_f32, k_f32, v_f32, x, wq, wo, k, v, q, ctx, acc,
          low_q, low_o, fields_q, fields_o, stream, plain, near_q, near_o, far_q, far_o,
          load_sem, send_sem, recv_sem, ready_sem):
    me = lax.axis_index("i")
    side = (me ^ 1, 3 - me)
    buffers = (low_q, low_o, fields_q, fields_o, stream, plain)
    barrier = pltpu.get_barrier_semaphore()

    loads = []

    def load(whole, *copies):
        sem = load_sem.at[len(loads)]
        for src, dst in copies:
            pltpu.make_async_copy(src, dst, sem).start()
        loads.append(pltpu.make_async_copy(whole, whole, sem))
        return loads[-1].wait

    def load_x(b):
        dst = x_f32.at[pl.ds(256 * b, 256)]
        return load(dst, (x_hbm.at[b], dst))

    def load_units(hbm, buf, group, batches=(0, 1)):
        if group in (0, 3):
            pairs = [(2 * (me ^ 2 if group else me), 2)]
        else:
            pairs = [(2 * chip + group - 1, 1) for chip in side]
        copies = [(hbm.at[2 * me + b, pl.ds(pl.multiple_of(128 * pair, 128), 128 * n)],
                   buf.at[pl.ds(128 * (4 * group + 2 * b + j), 128 * n)])
                  for b in batches for j, (pair, n) in enumerate(pairs)]
        return load(buf.at[pl.ds(512 * group + 256 * batches[0], 256 * len(batches))], *copies)

    def load_kv(group, batches=(0, 1)):
        return load_units(k_hbm, k_f32, group, batches), load_units(v_hbm, v_f32, group, batches)

    def copy(name, c, src, dst, target, rows=None):
        buf = _PARTS[name][0]
        rows = pl.ds(*(rows or _PARTS[name][1 + c]))
        return pltpu.make_async_remote_copy(
            buffers[buf].at[src, rows], buffers[buf].at[dst, rows],
            send_sem.at[buf + c if buf == _PLAIN else buf],
            recv_sem.at[2 * list(_PARTS).index(name) + c],
            device_id=(target,), device_id_type=_MESH)

    def outgoing(name, c):
        if name.startswith("far"):
            return copy(name, c, c, _FAR, side[1 - c])
        return copy(name, c, _OWN, c, side[c])

    def send(*names):
        for name in names:
            for c in range(2):
                outgoing(name, c).start()

    def wait(*names, sides=(0, 1)):
        for name in names:
            for c in sides:
                slot = _FAR if name.startswith("far") else c
                copy(name, c, slot, slot, me).wait_recv()

    def relay(when, arrived, onward):
        @pl.when(when)
        def _():
            wait(*arrived)
            send(onward)

    def wait_sent(*which):
        for buf in which:
            sent = buffers[buf].at[0:3, 0:_STREAM_ROWS] if buf == _STREAM else buffers[buf].at[0:3]
            pltpu.make_async_remote_copy(
                sent, sent, send_sem.at[buf], recv_sem.at[0],
                device_id=(me,), device_id_type=_MESH).wait_send()

    def signal_neighbours(sem):
        for chip in side:
            pl.semaphore_signal(sem, 1, device_id=(chip,), device_id_type=_MESH)

    def round_wq(h, start, size):
        w = _words(wq_f32[h, 32 * start:32 * (start + size), :]).reshape(size, 2, 8, 128)
        low_q[_OWN, pl.ds(16 * h + start, size)] = _fuse(w, _SIGN_MANTISSA)
        for r in range(start // 4, (start + size + 3) // 4):
            lo, hi = max(start, 4 * r), min(start + size, 4 * r + 4)
            wq[4 * h + r, 2 * (lo - 4 * r):2 * (hi - 4 * r)] = (
                w[lo - start:hi - start].reshape(-1, 8, 128))

    def round_wo(h):
        w = _words(wo_f32[:, 256 * h:256 * h + 256])
        for n in range(2):
            wo[pl.ds(4 * h + 2 * n, 2)] = w[:, 128 * n:128 * n + 128].reshape(2, 8, 8, 128)

    decoders = {}

    def decode(far, m, first, last):
        slots = (_FAR,) if far else (0, 1)
        senders = pl.ds(slots[0], len(slots))
        out = ((near_q, near_o), (far_q, far_o))[far][m]
        if far not in decoders:
            sent_plain = [stream[slot, _HEAD:_HEAD + 8][0, 0] == -1 for slot in slots]
            decoders[far] = sent_plain, _open_stream(stream.at[senders])
        sent_plain, state = decoders[far]
        for half in range(first // 4, (last + 3) // 4):
            top = _and(_move(_stream_row(stream.at[senders], _HEAD + m), -16 * half), 0xFFFF)
            state = _decode(top, (fields_q, fields_o)[m].at[senders], out,
                            max(first, 4 * half), min(last, 4 * half + 4), state)
        decoders[far] = sent_plain, state

        def use_plain(slot):
            if m == 0 and first == 0 and far:
                wait("far plain")
            elif m == 0 and first == 0:
                wait("plain", sides=(slot,))
                onward = outgoing("far plain", slot)
                onward.start()
                onward.wait_send()
            exponents = plain[slot, m, 4 * first:4 * last]
            out[slot % 2, 4 * first:4 * last, 0] = _or(exponents, _SIGN_MANTISSA)
            out[slot % 2, 4 * first:4 * last, 1] = _or(_rotl(exponents, 24), _SIGN_MANTISSA)

        @pl.when(sent_plain[0] | sent_plain[-1])
        def _():
            for slot, flag in zip(slots, sent_plain):
                pl.when(flag)(lambda: use_plain(slot))

    def round_x(b):
        x[128 * b:128 * b + 128] = _words(x_f32[256 * b:256 * b + 256] * _SCORE_SCALE)

    def round_k(*units):
        for u in units:
            k[128 * u:128 * u + 128] = pltpu.bitcast(k_f32[128 * u:128 * u + 128].astype(bf16).T, i32)

    def round_v(*units):
        for u in units:
            v[64 * u:64 * u + 64] = _words(v_f32[128 * u:128 * u + 128])

    def q_projection(group):
        if group == 0:
            pairs = [wq[4 * h:4 * h + 4].reshape(256, 128) for h in range(2)]
        else:
            pairs = [_rebuild(low_q[slot, 16 * h:16 * h + 16],
                              (far_q if slot == _FAR else near_q)[slot % 2, 16 * h:16 * h + 16])
                     for slot, h in _Q_GROUPS[group]]
        w = _halves(lax.concatenate(pairs, 1))

        def project(first, last):
            q[64 * first:64 * last, 256 * group:256 * group + 256] = _words(
                _dot(_halves(x[64 * first:64 * last]), w))

        return project

    def out_projection(group, first, last):
        if group == 0:
            tiles = [wo[2 * n:2 * n + 2].reshape(128, 128) for n in range(first, last)]
        else:
            tiles = [lax.concatenate(
                [_rebuild(low_o[slot, pl.ds(16 * h + 4 * n, 4)],
                          (far_o if slot == _FAR else near_o)[slot % 2, pl.ds(8 * n + 4 * h, 4)])
                 for slot, h in _O_GROUPS[group]], 0) for n in range(first, last)]
        w, cols = _halves(lax.concatenate(tiles, 1)), slice(128 * first, 128 * last)

        def project(*batches):
            for b in batches:
                rows = slice(256 * b, 256 * b + 256)
                r = _dot(_halves(ctx[128 * b:128 * b + 128, 256 * group:256 * group + 256]), w)
                if group > 0:
                    r = acc[rows, cols] + r
                if group < 3:
                    acc[rows, cols] = r
                else:
                    out_ref[rows, cols] = r.astype(out_ref.dtype)

        return project

    pending = {}

    def score(*units, tiles=(1, 0)):
        for u in units:
            b, col = u // 2 % 2, 256 * (u // 4) + 128 * (u % 2)
            for t in tiles:
                pending[u, t] = _scores(q[128 * b:128 * b + 128, col:col + 128], k, 128 * u, t)

    def store(*units, tiles=(1, 0)):
        for u in units:
            b, col = u // 2 % 2, 128 * _CONTEXT_COLUMN[2 * (u // 4) + u % 2]
            for t in tiles:
                ctx[pl.ds(128 * b + 64 * t, 64), col:col + 128] = _by_query(pending.pop((u, t)))

    def attend(*units, tiles=(1, 0), store_later=False):
        for u in units:
            for t in tiles:
                pending[u, t] = _context(pending[u, t], v, 64 * u, t)
                if not store_later:
                    store(u, tiles=(t,))

    wq_pieces = []
    for start, size in _FIRST_PIECES:
        dst = wq_f32.at[0, pl.ds(32 * start, 32 * size)]
        wq_pieces.append(load(dst, (wq_hbm.at[pl.ds(32 * start, 32 * size), pl.ds(0, 128)], dst)))
    pl.when(me != 2)(lambda: signal_neighbours(barrier))
    wq_rest = load(wq_f32.at[1], (wq_hbm.at[:, pl.ds(128, 128)], wq_f32.at[1]))
    wo_tiles = []
    for n in range(4):
        dst = wo_f32.at[:, pl.ds(128 * n, 128)]
        wo_tiles.append(load(dst, (wo_hbm.at[:, pl.ds(128 * n, 128)], dst)))
    odd, root, others = (me & 1) == 1, me == 0, me != 0
    pl.when(odd)(lambda: pl.semaphore_wait(barrier, 1))

    @pl.when(me == 2)
    def _():
        pl.semaphore_wait(barrier, 2)
        signal_neighbours(ready_sem)

    c = (me == 3).astype(i32)
    for arrived, rows in zip(wq_pieces, _FIRST_PIECES):
        arrived()
        round_wq(0, *rows)
        pl.when(others)(copy("q0", c, _OWN, c, jnp.where(me == 3, side[1], side[0]), rows).start)
        pl.when(me == 2)(copy("q0", 1, _OWN, 1, side[1], rows).start)
    x0, kv00, x1, kv01 = load_x(0), load_kv(0, (0,)), load_x(1), load_kv(0, (1,))

    zero = lax.full((8, 128), 0, i32)
    tops = [_choose_top(wq, 0)]
    code = _encode(wq, 0, tops[0], fields_q.at[_OWN], ((zero,) * _MAX_WORDS, zero, zero))
    wq_rest()
    round_wq(1, 0, 16)
    tops.append(_choose_top(wq, 1))
    code = _encode(wq, 1, tops[1], fields_q.at[_OWN], code)

    @pl.when(odd)
    def _():
        pl.semaphore_wait(ready_sem, 1)
        copy("q0", 1 - c, _OWN, 1 - c, jnp.where(me == 3, side[0], side[1]), (0, 16)).start()

    pl.when(others)(lambda: send("q fields", "q1 head"))
    for h in range(2):
        wo_tiles[2 * h]()
        wo_tiles[2 * h + 1]()
        round_wo(h)
        tops.append(_choose_top(wo, h))
        code = _encode(wo, h, tops[-1], fields_o.at[_OWN], code)
        if h == 0:
            @pl.when(root)
            def _():
                pl.semaphore_wait(barrier, 2)
                send("q0", "q fields", "q1 head")

    too_long = _write_stream(tops, code, stream.at[_OWN])
    for r in range(8):
        low_o[_OWN, pl.ds(16 * (r % 2) + 4 * (r // 2), 4)] = _fuse(
            wo[r].reshape(4, 2, 8, 128), _SIGN_MANTISSA)

    @pl.when(too_long)
    def _():
        stream[_OWN] = lax.full(stream.shape[1:], -1, i32)
        for m, ref in enumerate((wq, wo)):
            plain[_OWN, m] = _fuse(ref[...].reshape(32, 2, 8, 128), _EXPONENT)
        send("plain")
        for i in range(2):
            outgoing("plain", i).wait_send()

    send("stream", "q1 rest")
    kv1 = load_kv(1)
    x0()
    round_x(0)
    q_projection(0)(0, 2)
    kv00[0](), kv00[1]()
    round_k(0, 1)
    round_v(0, 1)
    score(0, tiles=(0,)), score(0, 1, tiles=(1,)), score(1, tiles=(0,))
    attend(0, tiles=(0,), store_later=True)
    attend(0, 1, tiles=(1,), store_later=True)
    attend(1, tiles=(0,), store_later=True)
    kv2 = load_kv(2)
    send("o fields 0", "o head")
    x1()
    round_x(1)
    q_projection(0)(2, 4)
    store(0, 1)
    wait("q0")
    send("far q0")
    kv01[0](), kv01[1]()
    round_k(2, 3)
    score(2, 3)
    out_projection(0, 0, 2)(0)
    round_v(2, 3)
    attend(2, 3)
    out_projection(0, 2, 4)(0)

    wait("q fields", "stream")
    send("far q fields", "far stream", "o fields 1")
    kv3 = load_kv(3)
    out_projection(0, 0, 4)(1)
    decode(False, 0, 0, 4)
    relay(others, ("q1 head", "q1 rest"), "far q1")
    send("o01")
    kv1[0]()
    q_projection(1)(0, 4)
    round_k(4, 5, 6, 7)
    decode(False, 0, 4, 8)
    relay(root, ("q1 head", "q1 rest"), "far q1")
    send("o2", "o3", "other o01")
    kv1[1](), kv2[0]()
    score(4, 5, 6)
    round_v(4, 5, 6, 7)
    project = q_projection(2)
    project(0, 1)
    attend(4)
    score(7)
    project(1, 2)
    attend(5, 6)
    round_k(8, 9, 10, 11)
    project(2, 3)
    attend(7)
    project(3, 4)
    relay(others, ("o fields 0", "o fields 1"), "far o fields")
    send("other o23")
    wait("far q fields", "far stream")
    kv2[1]()
    score(8, tiles=(0,)), score(8, 9, 10, 11, tiles=(1,)), score(9, 10, 11, tiles=(0,))
    round_v(8, 9, 10, 11)
    attend(8, tiles=(0,))
    attend(8, 9, 10, 11, tiles=(1,))
    attend(9, 10, 11, tiles=(0,), store_later=True)
    decode(True, 0, 0, 8)

    relay(others, ("o head", "o01"), "far o01")
    relay(root, ("o fields 0", "o fields 1"), "far o fields")
    wait("far q0", "far q1")
    kv3[0](), kv3[1]()
    q_projection(3)(0, 4)
    round_k(12, 13, 14, 15)
    store(9, 10, 11, tiles=(0,))
    decode(False, 1, 0, 6)
    relay(root, ("o head", "o01"), "far o01")
    wait("o2")
    send("far o2")
    relay(others, ("o3",), "far o3")
    score(12, 13, 14, 15)
    round_v(12, 13, 14, 15)
    project = out_projection(1, 0, 3)
    project(0)
    attend(12, 13)
    project(1)
    attend(14, 15, store_later=True)
    decode(False, 1, 6, 8)
    relay(root, ("o3",), "far o3")
    wait("other o01", "far o fields")
    out_projection(1, 3, 4)(0, 1)
    out_projection(2, 0, 2)(0, 1)
    store(14, 15)
    decode(True, 1, 0, 4)
    wait("other o23")
    out_projection(2, 2, 4)(0, 1)
    decode(True, 1, 4, 6)
    wait_sent(_LOW_Q, _FIELDS_Q, _FIELDS_O, _STREAM)
    wait("far o01")
    out_projection(3, 0, 2)(0, 1)
    decode(True, 1, 6, 8)
    wait("far o2")
    out_projection(3, 2, 3)(0, 1)
    wait("far o3")
    out_projection(3, 3, 4)(0, 1)
    wait_sent(_LOW_O)


def pallas_dist_sparse_attn_causalblk_htp_bs_b2_sq256_skv256_hq4_dh64_kernel(
    x: jax.Array,
    Wq: jax.Array,
    K_ext: jax.Array,
    V_ext: jax.Array,
    Wo: jax.Array,
):
    k_t = jnp.transpose(K_ext, (0, 2, 3, 1)).reshape(8, 1024, 256)
    v_t = jnp.transpose(V_ext, (0, 2, 3, 1)).reshape(8, 1024, 256)
    out = pl.pallas_call(
        _body,
        out_shape=jax.ShapeDtypeStruct((512, 512), bf16),
        in_specs=[pl.BlockSpec(memory_space=pltpu.HBM)] * 5,
        out_specs=pl.BlockSpec(memory_space=pltpu.VMEM),
        scratch_shapes=[
            pltpu.VMEM((512, 512), f32),
            pltpu.VMEM((2, 512, 128), f32),
            pltpu.VMEM((256, 512), f32),
            pltpu.VMEM((2048, 256), f32),
            pltpu.VMEM((2048, 256), f32),
            pltpu.VMEM((256, 512), i32),
            pltpu.VMEM((8, 8, 8, 128), i32),
            pltpu.VMEM((8, 8, 8, 128), i32),
            pltpu.VMEM((2048, 128), i32),
            pltpu.VMEM((1024, 256), i32),
            pltpu.VMEM((256, 1024), i32),
            pltpu.VMEM((256, 1024), i32),
            pltpu.VMEM((512, 512), f32),
            pltpu.VMEM((4, 32, 8, 128), i32),
            pltpu.VMEM((4, 32, 8, 128), i32),
            pltpu.VMEM((4, 8, 8, 128), i32),
            pltpu.VMEM((4, 8, 8, 128), i32),
            pltpu.VMEM((4, 56, 128), i32),
            pltpu.VMEM((4, 2, 32, 8, 128), i32),
            pltpu.VMEM((2, 32, 2, 8, 128), i32),
            pltpu.VMEM((2, 32, 2, 8, 128), i32),
            pltpu.VMEM((1, 32, 2, 8, 128), i32),
            pltpu.VMEM((1, 32, 2, 8, 128), i32),
            pltpu.SemaphoreType.DMA((20,)),
            pltpu.SemaphoreType.DMA((7,)),
            pltpu.SemaphoreType.DMA((2 * len(_PARTS),)),
            pltpu.SemaphoreType.REGULAR,
        ],
        compiler_params=pltpu.CompilerParams(
            collective_id=0,
            vmem_limit_bytes=48 << 20,
            flags={"XLA_TPU_FORCE_LP_LLO_SCHEDULER": True},
            disable_bounds_checks=True,
            disable_semaphore_checks=True,
        ),
    )(x, Wq, k_t, v_t, Wo)
    return out.reshape(x.shape)
```

```python
import jax
import jax.numpy as jnp
import numpy as np
from jax import lax
from jax.experimental import pallas as pl
from jax.experimental.pallas import tpu as pltpu

bf16, f32, i32 = jnp.bfloat16, jnp.float32, jnp.int32
_MESH = pl.DeviceIdType.MESH
_SCORE_SCALE = 0.125 * 1.4426950408889634


def _const(v):
    return np.uint32(v & 0xFFFFFFFF).astype(np.int32) if isinstance(v, int) else v


def _and(a, b):
    return lax.bitwise_and(a, _const(b))


def _or(a, b):
    return b if a is None else lax.bitwise_or(a, _const(b))


def _add(a, b):
    return b if a is None else lax.add(a, _const(b))


def _sub(a, b):
    return lax.sub(_const(a), _const(b))


def _shl(a, n):
    return lax.shift_left(_const(a), _const(n))


def _shr(a, n):
    return lax.shift_right_logical(_const(a), _const(n))


def _move(a, n):
    return a if n == 0 else (_shl(a, n) if n > 0 else _shr(a, -n))


def _rotl(a, n):
    return _or(_shl(a, n), _shr(a, 32 - n))


def _pick(mask, a, b):
    a, b = (lax.full(mask.shape, _const(v), i32) if isinstance(v, int) else v for v in (a, b))
    return lax.select(mask, a, b)


def _words(x):
    return pltpu.bitcast(x.astype(bf16), i32)


def _halves(w):
    return pltpu.bitcast(w, bf16)


_SIGN_MANTISSA = 0x807F807F
_EXPONENT = 0x7F807F80
_OWN_WORDS, _MAX_WORDS, _POOL_WORDS = 5, 9, 10
_HEAD = 8 * _OWN_WORDS
_POOL = _HEAD + 3
_STREAM_ROWS = _POOL + _POOL_WORDS


def _fuse(pairs, mask):
    return _or(_and(pairs[:, 0], mask), _rotl(_and(pairs[:, 1], mask), 8))


def _rebuild(low, coarse):
    out = []
    for k, bits in enumerate((low, _rotl(low, 24))):
        bits = _and(bits, _SIGN_MANTISSA)
        out.append(_or(_and(_sub(coarse[:, k], bits), _EXPONENT), bits))
    return lax.concatenate(out, 1).reshape(-1, 128)


def _choose_top(w_ref, half):
    peak = total = None
    for r in range(4 * half, 4 * half + 4):
        for j in (0, 4):
            w = w_ref[r, j:j + 4]
            m = lax.max(*(lax.bitcast_convert_type(_and(v, 0x3FFF8000), f32)
                          for v in (_shl(w, 15), _shr(w, 1))))
            peak = m if peak is None else lax.max(peak, m)
            total = _add(total, _and(_shr(w, 7), 0xFF00FF))
    peak = jnp.max(peak.reshape(32, 128), axis=0, keepdims=True)
    peak = _shr(lax.bitcast_convert_type(jnp.broadcast_to(peak, (8, 128)), i32), 15)
    total = _add(_and(total, 0xFFFF), _shr(total, 16)).reshape(32, 128).astype(f32)
    top = jnp.sum(total, axis=0, keepdims=True) * 0.25 + 469.0
    top = jnp.broadcast_to(top, (8, 128)).astype(i32)
    return _pick(lax.gt(peak, top), peak, top)


def _encode(w_ref, half, top, field_ref, stream):
    top = _or(_shl(top, 16), top)

    def run(r, stream):
        words, end, widest = stream
        fields = pos = b0 = b1 = None
        for j in range(8):
            gap = _sub(top, _and(w_ref[r, j], 0x7FFF7FFF))
            pair = None
            for depth, at in ((_and(_shr(gap, 7), 0x1FF), 2 * j), (_shr(gap, 23), 2 * j + 16)):
                deep = lax.gt(depth, _const(3))
                fields = _or(fields, _move(_pick(deep, 0, depth), at))
                n = _pick(deep, _sub(depth, _pick(lax.lt(depth, _const(7)), 3, 2)),
                          _pick(lax.eq(depth, _const(0)), 4, 0))
                pos, pair = _add(pos, n), _add(pair, n)
                stop, early = _shr(1 << 31, _and(pos, 31)), lax.lt(pos, _const(32))
                b0, b1 = _or(b0, _pick(early, stop, 0)), _or(b1, _pick(early, 0, stop))
            widest = _or(widest, pair)
        field_ref[r] = fields
        word, at = _shr(end, 5), _and(end, 31)
        back = _sub(31, at)
        parts = (_shr(b0, at), _or(_shr(b1, at), _shl(_add(b0, b0), back)), _shl(_add(b1, b1), back))
        here = [lax.eq(word, _const(i)) for i in range(_MAX_WORDS)]
        grown = []
        for i, w in enumerate(words):
            new = 0
            for k, part in enumerate(parts[:i + 1]):
                new = _pick(here[i - k], part, new)
            grown.append(_or(w, new))
        return tuple(grown), _add(end, pos), _or(widest, _shr(pos, 1))

    return lax.fori_loop(4 * half, 4 * half + 4, run, stream)


def _write_stream(tops, stream, ref):
    words, end, widest = stream
    extra = _sub(_shr(end, 5), _OWN_WORDS - 1)
    extra = _pick(lax.gt(extra, _const(0)), extra, 0)
    rows = [_add(lax.broadcasted_iota(i32, (8, 128), 0), 8 * i + _HEAD - _POOL) for i in range(2)]
    used = offsets = lax.full((8, 128), 0, i32)
    pool = [used, used]
    for s in range(8):
        offsets = _or(offsets, _move(_and(used, 15), 4 * s))
        ahead = [_sub(r, used) for r in rows]
        for k, word in enumerate(words[_OWN_WORDS:]):
            word = jnp.broadcast_to(word[s:s + 1], (8, 128))
            pool = [_pick(lax.eq(a, _const(k)), word, p) for a, p in zip(ahead, pool)]
        used = _add(used, jnp.broadcast_to(extra[s:s + 1], (8, 128)))
    heads = (_or(tops[0], _shl(tops[1], 16)), _or(tops[2], _shl(tops[3], 16)), offsets)
    for i, head in enumerate(heads):
        pool[0] = _pick(lax.eq(rows[0], _const(i + _HEAD - _POOL)), head, pool[0])
    over = (widest > 31) | (end >= 32 * _MAX_WORDS) | (used > _POOL_WORDS)
    over = jnp.max(jnp.where(over, 1.0, 0.0), axis=0, keepdims=True)
    over = jnp.broadcast_to(over, (8, 128)) > 0.0
    for i, w in enumerate(list(words[:_OWN_WORDS]) + pool):
        ref[8 * i:8 * i + 8] = _pick(over, -1, w)


def _too_long(stream_ref):
    return jnp.max(jnp.where(stream_ref[_HEAD:_HEAD + 1] == -1, 1.0, 0.0)) > 0.0


def _stream_row(stream_ref, i):
    return jnp.broadcast_to(stream_ref[:, i:i + 1, :], (stream_ref.shape[0], 8, 128))


def _open_stream(stream_ref):
    words = [stream_ref[:, 8 * i:8 * i + 8, :] for i in range(_OWN_WORDS)]
    sublane = lax.broadcasted_iota(i32, words[0].shape, 1)
    offset = _and(_shr(_stream_row(stream_ref, _HEAD + 2), _shl(sublane, 2)), 15)
    more = [-1] * (_MAX_WORDS - _OWN_WORDS)
    for i in range(_POOL_WORDS):
        mine = lax.eq(offset, _const(i))
        more = [_pick(mine, _stream_row(stream_ref, _POOL + i + k), m) if i + k < _POOL_WORDS else m
                for k, m in enumerate(more)]
    return tuple(words + more), lax.full(words[0].shape, 0, i32)


def _decode(top, field_ref, out_ref, first, last, state):
    base = _add(_or(_shl(top, 16), top), 0x80008000)

    def run(r, state):
        words, pos = state
        one, two = lax.gt(pos, _const(31)), lax.gt(pos, _const(63))
        words = words + (-1, -1)
        words = tuple(_pick(two, c, _pick(one, b, a)) for a, b, c in zip(words, words[1:], words[2:]))
        pos = _and(pos, 31)
        back = _sub(31, pos)
        w0, w1 = (_or(_shl(a, pos), _shr(_shr(b, 1), back)) for a, b in zip(words[:2], words[1:3]))
        fields = field_ref[:, r]
        for j in range(8):
            aligned, out, used = _move(fields, 7 - 2 * j), base, None
            for at in (7, 23):
                shallow = _and(aligned, 3 << at)
                escape = lax.eq(shallow, _const(0))
                w0 = _and(w0, 0x7FFFFFFF)
                n = _pick(escape, lax.clz(w0), 0)
                w0, used = _shl(w0, n), _add(used, n)
                deep = _shl(_add(n, _pick(lax.lt(n, _const(4)), 3, 2)), at)
                out = _sub(out, _pick(lax.bitwise_and(escape, lax.ne(n, _const(4))), deep, shallow))
            if j < 7:
                w0, w1 = _or(w0, _shr(_shr(w1, 1), _sub(31, used))), _shl(w1, used)
            pos = _add(pos, used)
            out_ref[:, 4 * r + j // 2, j % 2] = out
        return words, pos

    return lax.fori_loop(first, last, run, state, unroll=True)


def _dot(a, b):
    return jnp.dot(a, b, preferred_element_type=f32)


def _low_lanes(rows):
    return lax.broadcasted_iota(i32, (rows, 128), 1) < 64


def _scores(q, k_ref, row, tile):
    low, out = _low_lanes(32), [None, None]
    for j in (1, 0):
        block = 2 * tile + j
        qq = q[32 * block:32 * block + 32]
        heads = [_pick(low, qq, 0), _pick(low, 0, qq)]
        out[j] = lax.dot_general(
            _halves(k_ref[row:row + 32 * (block + 1), :]),
            _halves(lax.concatenate(heads[::1 - 2 * j], 0)),
            (((1,), (1,)), ((), ())), preferred_element_type=f32)
    return out


def _context(scores, v_ref, row, tile):
    keys = 128 * (tile + 1)
    p, inv = [], []
    for s in scores:
        p.append(lax.exp2(s - jnp.max(s, axis=0, keepdims=True)))
        inv.append(1.0 / jnp.sum(p[-1], axis=0, keepdims=True))
    p[0] = lax.concatenate([p[0], lax.full((64, 128), 0.0, f32)], 0)
    low, low_row = _low_lanes(keys), _low_lanes(1)
    heads = [(lax.select(low, p[h], p[1 - h]).astype(bf16), lax.select(low_row, inv[h], inv[1 - h]))
             for h in range(2)]
    return lax.concatenate(
        [_dot(_halves(v_ref[row + 32 * h:row + 32 * h + 32, 0:keys]), weights) * scale
         for h, (weights, scale) in enumerate(heads)], 0)


def _by_query(context):
    c, low = pltpu.bitcast(context.astype(bf16).T, i32), _low_lanes(32)
    return lax.concatenate([_pick(low, c[0:32], c[32:64]), _pick(low, c[32:64], c[0:32])], 0)


_FAR, _OWN = 2, 3
_LOW_Q, _LOW_O, _FIELDS_Q, _FIELDS_O, _STREAM, _PLAIN = range(6)
_PARTS = {
    "q0": (_LOW_Q, (0, 16), (0, 16)),
    "q1": (_LOW_Q, (16, 8), (24, 8)),
    "other q1": (_LOW_Q, (24, 8), (16, 8)),
    "far q0": (_LOW_Q, (0, 8), (8, 8)),
    "far q1": (_LOW_Q, (16, 8), (24, 8)),
    "q fields": (_FIELDS_Q, (0, 8), (0, 8)),
    "far q fields": (_FIELDS_Q, (0, 4), (4, 4)),
    "o0 fields": (_FIELDS_O, (0, 2), (0, 2)),
    "o12 fields": (_FIELDS_O, (2, 4), (2, 4)),
    "o3 fields": (_FIELDS_O, (6, 2), (6, 2)),
    "far o0 fields": (_FIELDS_O, (0, 1), (1, 1)),
    "far o12 fields": (_FIELDS_O, (2, 2), (4, 2)),
    "far o3 fields": (_FIELDS_O, (6, 1), (7, 1)),
    "stream": (_STREAM, (0, _STREAM_ROWS), (0, _STREAM_ROWS)),
    "far stream": (_STREAM, (0, 24), (24, _STREAM_ROWS - 24)),
    "o0": (_LOW_O, (0, 4), (16, 4)),
    "o1": (_LOW_O, (4, 4), (20, 4)),
    "o2": (_LOW_O, (8, 4), (24, 4)),
    "o3": (_LOW_O, (12, 4), (28, 4)),
    "other o012": (_LOW_O, (16, 12), (0, 12)),
    "other o3": (_LOW_O, (28, 4), (12, 4)),
    "far o0": (_LOW_O, (0, 4), (16, 4)),
    "far o1": (_LOW_O, (4, 4), (20, 4)),
    "far o2": (_LOW_O, (8, 4), (24, 4)),
    "far o3": (_LOW_O, (12, 4), (28, 4)),
    "plain": (_PLAIN, (0, 2), (0, 2)),
    "far plain": (_PLAIN, (0, 1), (1, 1)),
}
_FIRST_PIECES = ((0, 2), (2, 6), (8, 8))
_Q_GROUPS = (None, ((0, 0), (1, 0)), ((0, 1), (1, 1)), ((_FAR, 0), (_FAR, 1)))
_O_GROUPS = (None, ((0, 0), (1, 1)), ((0, 1), (1, 0)), ((_FAR, 0), (_FAR, 1)))
_CONTEXT_COLUMN = (0, 1, 2, 5, 4, 3, 6, 7)


def _body(x_hbm, wq_hbm, k_hbm, v_hbm, wo_hbm, out_ref,
          x_f32, wq_f32, wo_f32, k_f32, v_f32, x, wq, wo, k, v, q, ctx, acc,
          low_q, low_o, fields_q, fields_o, stream, plain, near_q, near_o, far_q, far_o,
          load_sem, send_sem, recv_sem, ready_sem):
    me = lax.axis_index("i")
    side = (me ^ 1, 3 - me)
    buffers = (low_q, low_o, fields_q, fields_o, stream, plain)
    barrier = pltpu.get_barrier_semaphore()

    loads = []

    def load(whole, *copies):
        sem = load_sem.at[len(loads)]
        for src, dst in copies:
            pltpu.make_async_copy(src, dst, sem).start()
        loads.append(pltpu.make_async_copy(whole, whole, sem))
        return loads[-1].wait

    def load_x(b):
        dst = x_f32.at[pl.ds(256 * b, 256)]
        return load(dst, (x_hbm.at[b], dst))

    def load_units(hbm, buf, group, batches=(0, 1)):
        if group in (0, 3):
            pairs = [(2 * (me ^ 2 if group else me), 2)]
        else:
            pairs = [(2 * chip + group - 1, 1) for chip in side]
        copies = [(hbm.at[2 * me + b, pl.ds(pl.multiple_of(128 * pair, 128), 128 * n)],
                   buf.at[pl.ds(128 * (4 * group + 2 * b + j), 128 * n)])
                  for b in batches for j, (pair, n) in enumerate(pairs)]
        return load(buf.at[pl.ds(512 * group + 256 * batches[0], 256 * len(batches))], *copies)

    def load_kv(group, batches=(0, 1)):
        return load_units(k_hbm, k_f32, group, batches), load_units(v_hbm, v_f32, group, batches)

    def copy(name, c, src, dst, target, rows=None):
        buf = _PARTS[name][0]
        rows = pl.ds(*(rows or _PARTS[name][1 + c]))
        return pltpu.make_async_remote_copy(
            buffers[buf].at[src, rows], buffers[buf].at[dst, rows],
            send_sem.at[buf + c + 2 * name.startswith("far") if buf == _PLAIN else buf],
            recv_sem.at[2 * list(_PARTS).index(name) + c],
            device_id=(target,), device_id_type=_MESH)

    def outgoing(name, c):
        if name.startswith("far"):
            return copy(name, c, c, _FAR, side[1 - c])
        return copy(name, c, _OWN, c, side[c])

    def send(*names):
        for name in names:
            for c in range(2):
                outgoing(name, c).start()

    def wait(*names, sides=(0, 1)):
        for name in names:
            for c in sides:
                slot = _FAR if name.startswith("far") else c
                copy(name, c, slot, slot, me).wait_recv()

    def relay(when, arrived, onward):
        @pl.when(when)
        def _():
            wait(*arrived)
            send(onward)

    def wait_sent(*which):
        for buf in which:
            sent = buffers[buf].at[0:3, 0:_STREAM_ROWS] if buf == _STREAM else buffers[buf].at[0:3]
            pltpu.make_async_remote_copy(
                sent, sent, send_sem.at[buf], recv_sem.at[0],
                device_id=(me,), device_id_type=_MESH).wait_send()

    def signal_neighbours(sem):
        for chip in side:
            pl.semaphore_signal(sem, 1, device_id=(chip,), device_id_type=_MESH)

    def round_wq(h, start, size):
        w = _words(wq_f32[h, 32 * start:32 * (start + size), :]).reshape(size, 2, 8, 128)
        low_q[_OWN, pl.ds(16 * h + start, size)] = _fuse(w, _SIGN_MANTISSA)
        for r in range(start // 4, (start + size + 3) // 4):
            lo, hi = max(start, 4 * r), min(start + size, 4 * r + 4)
            wq[4 * h + r, 2 * (lo - 4 * r):2 * (hi - 4 * r)] = (
                w[lo - start:hi - start].reshape(-1, 8, 128))

    def round_wo(h):
        w = _words(wo_f32[:, 256 * h:256 * h + 256])
        for n in range(2):
            wo[pl.ds(4 * h + 2 * n, 2)] = w[:, 128 * n:128 * n + 128].reshape(2, 8, 8, 128)

    decoders = {}

    def decode(far, m, first, last):
        slots = (_FAR,) if far else (0, 1)
        senders = pl.ds(slots[0], len(slots))
        out = ((near_q, near_o), (far_q, far_o))[far][m]
        if far not in decoders:
            sent_plain = [_too_long(stream.at[slot]) for slot in slots]
            decoders[far] = sent_plain, _open_stream(stream.at[senders])
        sent_plain, state = decoders[far]
        for half in range(first // 4, (last + 3) // 4):
            top = _and(_move(_stream_row(stream.at[senders], _HEAD + m), -16 * half), 0xFFFF)
            state = _decode(top, (fields_q, fields_o)[m].at[senders], out,
                            max(first, 4 * half), min(last, 4 * half + 4), state)
        decoders[far] = sent_plain, state

        def use_plain(slot):
            if m == 0 and first == 0 and far:
                wait("far plain")
            elif m == 0 and first == 0:
                wait("plain", sides=(slot,))
                outgoing("far plain", slot).start()
            elif m == 1 and last == 8 and not far:
                outgoing("far plain", slot).wait_send()
            exponents = plain[slot, m, 4 * first:4 * last]
            out[slot % 2, 4 * first:4 * last, 0] = _or(exponents, _SIGN_MANTISSA)
            out[slot % 2, 4 * first:4 * last, 1] = _or(_rotl(exponents, 24), _SIGN_MANTISSA)

        @pl.when(sent_plain[0] | sent_plain[-1])
        def _():
            for slot, flag in zip(slots, sent_plain):
                pl.when(flag)(lambda: use_plain(slot))

    def round_x(b):
        x[128 * b:128 * b + 128] = _words(x_f32[256 * b:256 * b + 256] * _SCORE_SCALE)

    def round_k(*units):
        for u in units:
            k[128 * u:128 * u + 128] = pltpu.bitcast(k_f32[128 * u:128 * u + 128].astype(bf16).T, i32)

    def round_v(*units):
        for u in units:
            v[64 * u:64 * u + 64] = _words(v_f32[128 * u:128 * u + 128])

    def q_projection(group):
        if group == 0:
            pairs = [wq[4 * h:4 * h + 4].reshape(256, 128) for h in range(2)]
        else:
            pairs = [_rebuild(low_q[slot, 16 * h:16 * h + 16],
                              (far_q if slot == _FAR else near_q)[slot % 2, 16 * h:16 * h + 16])
                     for slot, h in _Q_GROUPS[group]]
        w = _halves(lax.concatenate(pairs, 1))

        def project(first, last):
            q[64 * first:64 * last, 256 * group:256 * group + 256] = _words(
                _dot(_halves(x[64 * first:64 * last]), w))

        return project

    def out_projection(group, first, last):
        if group == 0:
            tiles = [wo[2 * n:2 * n + 2].reshape(128, 128) for n in range(first, last)]
        else:
            tiles = [lax.concatenate(
                [_rebuild(low_o[slot, pl.ds(16 * h + 4 * n, 4)],
                          (far_o if slot == _FAR else near_o)[slot % 2, pl.ds(8 * n + 4 * h, 4)])
                 for slot, h in _O_GROUPS[group]], 0) for n in range(first, last)]
        w, cols = _halves(lax.concatenate(tiles, 1)), slice(128 * first, 128 * last)

        def project(*batches):
            for b in batches:
                rows = slice(256 * b, 256 * b + 256)
                r = _dot(_halves(ctx[128 * b:128 * b + 128, 256 * group:256 * group + 256]), w)
                if group > 0:
                    r = acc[rows, cols] + r
                if group < 3:
                    acc[rows, cols] = r
                else:
                    out_ref[rows, cols] = r.astype(out_ref.dtype)

        return project

    pending = {}

    def score(*units, tiles=(1, 0)):
        for u in units:
            b, col = u // 2 % 2, 256 * (u // 4) + 128 * (u % 2)
            for t in tiles:
                pending[u, t] = _scores(q[128 * b:128 * b + 128, col:col + 128], k, 128 * u, t)

    def store(*units, tiles=(1, 0)):
        for u in units:
            b, col = u // 2 % 2, 128 * _CONTEXT_COLUMN[2 * (u // 4) + u % 2]
            for t in tiles:
                ctx[pl.ds(128 * b + 64 * t, 64), col:col + 128] = _by_query(pending.pop((u, t)))

    def attend(*units, tiles=(1, 0), store_later=False):
        for u in units:
            for t in tiles:
                pending[u, t] = _context(pending[u, t], v, 64 * u, t)
                if not store_later:
                    store(u, tiles=(t,))

    wq_pieces = []
    for start, size in _FIRST_PIECES:
        dst = wq_f32.at[0, pl.ds(32 * start, 32 * size)]
        wq_pieces.append(load(dst, (wq_hbm.at[pl.ds(32 * start, 32 * size), pl.ds(0, 128)], dst)))
    pl.when(me != 2)(lambda: signal_neighbours(barrier))
    wq_rest = load(wq_f32.at[1], (wq_hbm.at[:, pl.ds(128, 128)], wq_f32.at[1]))
    wo_tiles = []
    for n in range(4):
        dst = wo_f32.at[:, pl.ds(128 * n, 128)]
        wo_tiles.append(load(dst, (wo_hbm.at[:, pl.ds(128 * n, 128)], dst)))
    odd, root, others = (me & 1) == 1, me == 0, me != 0
    pl.when(odd)(lambda: pl.semaphore_wait(barrier, 1))

    @pl.when(me == 2)
    def _():
        pl.semaphore_wait(barrier, 2)
        signal_neighbours(ready_sem)

    c = (me == 3).astype(i32)
    for arrived, rows in zip(wq_pieces, _FIRST_PIECES):
        arrived()
        round_wq(0, *rows)
        pl.when(others)(copy("q0", c, _OWN, c, jnp.where(me == 3, side[1], side[0]), rows).start)
        pl.when(me == 2)(copy("q0", 1, _OWN, 1, side[1], rows).start)
    x0, kv00, x1, kv01 = load_x(0), load_kv(0, (0,)), load_x(1), load_kv(0, (1,))

    zero = lax.full((8, 128), 0, i32)
    tops = [_choose_top(wq, 0)]
    code = _encode(wq, 0, tops[0], fields_q.at[_OWN], ((zero,) * _MAX_WORDS, zero, zero))
    wq_rest()
    round_wq(1, 0, 16)
    tops.append(_choose_top(wq, 1))
    code = _encode(wq, 1, tops[1], fields_q.at[_OWN], code)

    @pl.when(odd)
    def _():
        pl.semaphore_wait(ready_sem, 1)
        copy("q0", 1 - c, _OWN, 1 - c, jnp.where(me == 3, side[0], side[1]), (0, 16)).start()

    pl.when(others)(lambda: send("q fields"))
    for h in range(2):
        wo_tiles[2 * h]()
        wo_tiles[2 * h + 1]()
        round_wo(h)
        tops.append(_choose_top(wo, h))
        code = _encode(wo, h, tops[-1], fields_o.at[_OWN], code)
        if h == 0:
            @pl.when(root)
            def _():
                pl.semaphore_wait(barrier, 2)
                send("q0", "q fields")

    _write_stream(tops, code, stream.at[_OWN])
    send("stream", "q1", "other q1")
    too_long = _too_long(stream.at[_OWN])
    for r in range(8):
        low_o[_OWN, pl.ds(16 * (r % 2) + 4 * (r // 2), 4)] = _fuse(
            wo[r].reshape(4, 2, 8, 128), _SIGN_MANTISSA)

    @pl.when(too_long)
    def _():
        for m, ref in enumerate((wq, wo)):
            plain[_OWN, m] = _fuse(ref[...].reshape(32, 2, 8, 128), _EXPONENT)
        send("plain")

    kv1 = load_kv(1)
    x0()
    round_x(0)
    q_projection(0)(0, 2)
    kv00[0]()
    kv00[1]()
    round_k(0, 1)
    round_v(0, 1)
    score(0, tiles=(0,))
    score(0, 1, tiles=(1,))
    score(1, tiles=(0,))
    attend(0, tiles=(0,), store_later=True)
    attend(0, 1, tiles=(1,), store_later=True)
    attend(1, tiles=(0,), store_later=True)
    kv2 = load_kv(2)
    send("o0 fields", "o0")
    x1()
    round_x(1)
    q_projection(0)(2, 4)
    store(0, 1)
    wait("q0")
    send("far q0")
    kv01[0]()
    round_k(2, 3)
    kv01[1]()
    score(2, tiles=(0,))
    score(2, 3, tiles=(1,))
    score(3, tiles=(0,))
    round_v(2, 3)
    attend(2, tiles=(0,))
    out_projection(0, 0, 2)(0)
    attend(2, 3, tiles=(1,))
    attend(3, tiles=(0,))
    out_projection(0, 2, 4)(0)

    wait("q fields", "stream")
    send("far q fields", "far stream", "o12 fields")
    kv3 = load_kv(3)
    out_projection(0, 0, 4)(1)
    decode(False, 0, 0, 4)
    wait("q1")
    send("far q1", "o1", "o3 fields", "o2")
    kv1[0]()
    q_projection(1)(0, 4)
    round_k(4, 5, 6, 7)
    decode(False, 0, 4, 8)
    send("o3", "other o012")
    wait("other q1")
    kv1[1]()
    kv2[0]()
    score(4, 5, 6)
    round_v(4, 5, 6, 7)
    project = q_projection(2)
    project(0, 1)
    attend(4)
    score(7)
    project(1, 2)
    attend(5, 6)
    round_k(8, 9, 10, 11)
    project(2, 3)
    attend(7)
    project(3, 4)
    wait("o0 fields")
    send("far o0 fields", "other o3")
    wait("far q fields", "far stream")
    kv2[1]()
    score(8, tiles=(0,))
    score(8, 9, 10, 11, tiles=(1,))
    round_v(8, 9, 10, 11)
    attend(8, tiles=(0,))
    score(9, tiles=(0,))
    attend(8, tiles=(1,))
    score(10, tiles=(0,))
    attend(9, tiles=(1,))
    score(11, tiles=(0,))
    attend(10, 11, tiles=(1,))
    attend(9, 10, 11, tiles=(0,), store_later=True)
    decode(True, 0, 0, 8)

    wait("o12 fields", "o0")
    send("far o12 fields", "far o0")
    relay(others, ("o1",), "far o1")
    wait("far q0", "far q1")
    kv3[0]()
    kv3[1]()
    q_projection(3)(0, 4)
    round_k(12, 13, 14, 15)
    store(9, 10, 11, tiles=(0,))
    decode(False, 1, 0, 6)
    relay(root, ("o1",), "far o1")
    wait("o3 fields", "o2")
    send("far o3 fields", "far o2")
    relay(others, ("o3",), "far o3")
    score(12, tiles=(0,))
    score(12, 13, 14, 15, tiles=(1,))
    score(13, 14, tiles=(0,))
    round_v(12, 13, 14, 15)
    project = out_projection(1, 0, 2)
    project(0)
    attend(12, tiles=(0,))
    score(15, tiles=(0,))
    attend(12, tiles=(1,))
    project(1)
    attend(13, 14, 15, tiles=(1,))
    attend(13, tiles=(0,))
    attend(14, tiles=(0,), store_later=True)
    out_projection(1, 2, 3)(0, 1)
    attend(15, tiles=(0,), store_later=True)
    decode(False, 1, 6, 8)
    relay(root, ("o3",), "far o3")
    wait("other o012", "far o0 fields")
    out_projection(1, 3, 4)(0, 1)
    out_projection(2, 0, 3)(0, 1)
    store(14, 15, tiles=(0,))
    decode(True, 1, 0, 2)

    @pl.when(too_long)
    def _():
        for i in range(2):
            outgoing("plain", i).wait_send()

    wait("other o3", "far o12 fields", "far o0")
    out_projection(2, 3, 4)(0, 1)
    out_projection(3, 0, 1)(0, 1)
    decode(True, 1, 2, 6)
    wait("far o3 fields", "far o1")
    out_projection(3, 1, 2)(0, 1)
    decode(True, 1, 6, 8)
    wait("far o2")
    out_projection(3, 2, 3)(0, 1)
    wait_sent(_LOW_Q, _FIELDS_Q, _FIELDS_O, _STREAM)
    wait("far o3")
    out_projection(3, 3, 4)(0, 1)
    wait_sent(_LOW_O)


def pallas_dist_sparse_attn_causalblk_htp_bs_b2_sq256_skv256_hq4_dh64_kernel(
    x: jax.Array,
    Wq: jax.Array,
    K_ext: jax.Array,
    V_ext: jax.Array,
    Wo: jax.Array,
):
    k_t = jnp.transpose(K_ext, (0, 2, 3, 1)).reshape(8, 1024, 256)
    v_t = jnp.transpose(V_ext, (0, 2, 3, 1)).reshape(8, 1024, 256)
    out = pl.pallas_call(
        _body,
        out_shape=jax.ShapeDtypeStruct((512, 512), bf16),
        in_specs=[pl.BlockSpec(memory_space=pltpu.HBM)] * 5,
        out_specs=pl.BlockSpec(memory_space=pltpu.VMEM),
        scratch_shapes=[
            pltpu.VMEM((512, 512), f32),
            pltpu.VMEM((2, 512, 128), f32),
            pltpu.VMEM((256, 512), f32),
            pltpu.VMEM((2048, 256), f32),
            pltpu.VMEM((2048, 256), f32),
            pltpu.VMEM((256, 512), i32),
            pltpu.VMEM((8, 8, 8, 128), i32),
            pltpu.VMEM((8, 8, 8, 128), i32),
            pltpu.VMEM((2048, 128), i32),
            pltpu.VMEM((1024, 256), i32),
            pltpu.VMEM((256, 1024), i32),
            pltpu.VMEM((256, 1024), i32),
            pltpu.VMEM((512, 512), f32),
            pltpu.VMEM((4, 32, 8, 128), i32),
            pltpu.VMEM((4, 32, 8, 128), i32),
            pltpu.VMEM((4, 8, 8, 128), i32),
            pltpu.VMEM((4, 8, 8, 128), i32),
            pltpu.VMEM((4, 56, 128), i32),
            pltpu.VMEM((4, 2, 32, 8, 128), i32),
            pltpu.VMEM((2, 32, 2, 8, 128), i32),
            pltpu.VMEM((2, 32, 2, 8, 128), i32),
            pltpu.VMEM((1, 32, 2, 8, 128), i32),
            pltpu.VMEM((1, 32, 2, 8, 128), i32),
            pltpu.SemaphoreType.DMA((20,)),
            pltpu.SemaphoreType.DMA((9,)),
            pltpu.SemaphoreType.DMA((2 * len(_PARTS),)),
            pltpu.SemaphoreType.REGULAR,
        ],
        compiler_params=pltpu.CompilerParams(
            collective_id=0,
            vmem_limit_bytes=48 << 20,
            flags={"XLA_TPU_FORCE_LP_LLO_SCHEDULER": True},
            disable_bounds_checks=True,
            disable_semaphore_checks=True,
        ),
    )(x, Wq, k_t, v_t, Wo)
    return out.reshape(x.shape)
```
